```python
import numpy as np

kernel_name = "dist_sparse_attn_strided_kvseq_b1_sq256_skv4096_hq8_dh128"

def setup_inputs():
    x = np.random.randn(1, 256, 1024).astype(np.float32)
    Wq = np.random.randn(1024, 1024).astype(np.float32) * 0.02
    K_ext = np.random.randn(1, 16384, 8, 128).astype(np.float32)
    V_ext = np.random.randn(1, 16384, 8, 128).astype(np.float32)
    Wo = np.random.randn(1024, 1024).astype(np.float32) * 0.02
    return {"x": x, "Wq": Wq, "K_ext": K_ext, "V_ext": V_ext, "Wo": Wo}

def reference(x, Wq, K_ext, V_ext, Wo):
    B, Sq, Skv, Hq, Dh = 1, 256, 16384, 8, 128
    Q = (x @ Wq).reshape(B, Sq, Hq, Dh)
    qb = (np.arange(Sq) // 64)[:, None]
    kb = (np.arange(Skv) // 64)[None, :]
    mask = (qb == kb) | ((kb % 4) == (qb % 4))
    scores = np.einsum('bihd,bjhd->bhij', Q, K_ext).astype(np.float32) * 0.08838834764831843
    scores = np.where(mask[None, None, :, :], scores, -1e9)
    scores_max = scores.max(axis=-1, keepdims=True)
    w = np.exp(scores - scores_max)
    row_keep = mask.any(axis=1)
    w_sum = np.where(row_keep[None, None, :, None], w.sum(axis=-1, keepdims=True), 1.0)
    w = w / w_sum
    w = np.where(row_keep[None, None, :, None], w, 0.0)
    ctx = np.einsum('bhij,bjhd->bihd', w, V_ext).reshape(B, Sq, Hq * Dh)
    return ctx @ Wo
```

```python
import jax
import jax.numpy as jnp
from jax import lax
from jax.experimental import pallas as pl
from jax.experimental.pallas import tpu as pltpu

NC = 4
QB = 64
NH = 8
DH = 128
DM = 1024
NG = 16
NBH = 5
NTH = NH - NBH
NBU = NC * NBH
NTU = NC * NTH
NU = NBU + NTU
TAIL_LAG = 2
VP = 2
Q_SCALE = 0.08838834764831843 * 1.4426950408889634

F32 = jnp.float32
BF16 = jnp.bfloat16
MESH = pl.DeviceIdType.MESH
NT_DIMS = (((1,), (1,)), ((), ()))

UNITS = [(c, h) for c in range(NC) for h in range(NBH)] + [
    (c, h) for h in range(NBH, NH) for c in range(NC)
]


def _body(
    x_hbm, wq_hbm, k_hbm, v_hbm, wo_hbm, out_ref,
    kbuf, vbuf, xf, xb, wqf, wqb, wof, wob, qb, po,
    ls, bo, bs, lts, to, ts, ct, ob,
    ksem, vsem, vpsem, xlsem, wlsem, wtsem,
    xs_s, xs_r, q_s, q_r, bo_s, bo_r, bs_s, bs_r,
    ob_s, ob_r, to_s, to_r, ts_s, ts_r,
):
    me = lax.axis_index("i")
    half = me // 2
    is_qmaker = me % 2 == 1

    def remote(src, dst, ssem, rsem, dev):
        return pltpu.make_async_remote_copy(
            src, dst, ssem, rsem, device_id=(dev,), device_id_type=MESH)

    def wait_all(buf, sem):
        pltpu.make_async_copy(buf, buf, sem).wait()

    gp = NG // VP

    def issue_units(lo, hi):
        for u in range(lo, hi):
            c, h = UNITS[u]
            pltpu.make_async_copy(
                k_hbm.at[:, c, :, h, :], kbuf.at[u], ksem.at[u]).start()
            if u < NU - 1:
                pltpu.make_async_copy(
                    v_hbm.at[:, c, :, h, :], vbuf.at[u], vsem.at[u]).start()
            else:
                for p in range(VP):
                    pltpu.make_async_copy(
                        v_hbm.at[pl.ds(p * gp, gp), c, :, h, :],
                        vbuf.at[u, pl.ds(p * gp, gp)], vpsem.at[p]).start()

    def x_load(c):
        return pltpu.make_async_copy(
            x_hbm.at[0, pl.ds(c * QB, QB), :], xf.at[c], xlsem.at[c])

    def wq_load(hf):
        return pltpu.make_async_copy(
            wq_hbm.at[:, pl.ds(hf * 512, 512)], wqf, wlsem)

    def wo_bulk_load():
        rows = pl.ds(0, NBH * DH)
        return pltpu.make_async_copy(wo_hbm.at[rows], wof.at[rows], wlsem)

    def wo_tail_load(i):
        rows = pl.ds((NBH + i) * DH, DH)
        return pltpu.make_async_copy(
            wo_hbm.at[rows], wof.at[rows], wtsem.at[i])

    @pl.when(me == 2)
    def _():
        for c in range(NC):
            x_load(c).start()

    @pl.when(me == 1)
    def _():
        wq_load(0).start()

    @pl.when(me == 3)
    def _():
        wq_load(1).start()

    @pl.when(me == 0)
    def _():
        wo_bulk_load().start()

    issue_units(0, 2 * NBH)

    barrier = pltpu.get_barrier_semaphore()
    for d in (1, 2, 3):
        pl.semaphore_signal(
            barrier, 1, device_id=((me + d) % 4,), device_id_type=MESH)
    pl.semaphore_wait(barrier, 3)

    def x_send(c, k):
        return remote(xb.at[c], xb.at[c], xs_s.at[c, k], xs_r.at[c], 1 + 2 * k)

    def q_send(c, k):
        rows = qb.at[c, pl.ds(half * 4, 4)]
        dev = (0, 2, 4 - me)[k]
        return remote(rows, rows, q_s.at[c, k], q_r.at[c, half], dev)

    @pl.when(me == 2)
    def _():
        for c in range(NC):
            x_load(c).wait()
            xb[c] = xf[c].astype(BF16)
            x_send(c, 0).start()
            x_send(c, 1).start()

    @pl.when(is_qmaker)
    def _():
        wq_load(0).wait()
        wqb[...] = wqf[...].astype(BF16)
        for c in range(NC):
            wait_all(xb.at[c], xs_r.at[c])
            q = jnp.dot(xb[c], wqb[...], preferred_element_type=F32) * Q_SCALE
            for i in range(4):
                qb[c, half * 4 + i] = q[:, i * DH:(i + 1) * DH].astype(BF16)
            for k in range(3):
                q_send(c, k).start()
            if c == 1:
                issue_units(2 * NBH, 3 * NBH)

    @pl.when(me == 0)
    def _():
        wo_bulk_load().wait()
        wob[0:NBH * DH, :] = wof[0:NBH * DH, :].astype(BF16)

    eye = (lax.broadcasted_iota(jnp.int32, (QB, DH), 0)
           == lax.broadcasted_iota(jnp.int32, (QB, DH), 1))
    sub8 = lax.broadcasted_iota(jnp.int32, (8, DH), 0)

    def to_row(col):
        return jnp.sum(jnp.where(eye, col, 0.0), axis=0, keepdims=True)

    def to_col(row):
        return jnp.sum(jnp.where(eye, row, 0.0), axis=1, keepdims=True)

    def scores(u, c, h):
        k = kbuf[u].reshape(NG * QB, DH).astype(BF16)
        s = lax.dot_general(qb[c, h], k, NT_DIMS, preferred_element_type=F32)
        m = jnp.max(s, axis=1, keepdims=True)
        p = jnp.exp2(s - m)
        l = jnp.sum(p, axis=1, keepdims=True)
        return p.astype(BF16), 1.0 / l, m + jnp.log2(l)

    def merge_weights(stats):
        m = jnp.maximum(jnp.maximum(stats[0], stats[1]),
                        jnp.maximum(stats[2], stats[3]))
        e = [jnp.exp2(s - m) for s in stats]
        inv = 1.0 / (e[0] + e[1] + e[2] + e[3])
        return [x * inv for x in e]

    def bo_send(c, h):
        u = c * NBH + h
        return remote(po.at[u], bo.at[c, me - 1, h], bo_s.at[u], bo_r.at[c], 0)

    def bs_send(c):
        return remote(ls.at[c], bs.at[c, me - 1], bs_s.at[c], bs_r.at[c], 0)

    def ob_send(c, k):
        dev = (1, 3, 2)[k]
        return remote(ob.at[c], ob.at[c], ob_s.at[c, k], ob_r.at[c], dev)

    def project_bulk(c):
        @pl.when(me == 0)
        def _():
            wait_all(bs.at[c], bs_r.at[c])
            wait_all(bo.at[c], bo_r.at[c])
            w = merge_weights([ls[c]] + [bs[c, j] for j in range(3)])
            ctx = []
            for h in range(NBH):
                acc = to_col(w[0][h:h + 1]) * po[c * NBH + h].astype(F32)
                for j in range(3):
                    acc += to_col(w[j + 1][h:h + 1]) * bo[c, j, h].astype(F32)
                ctx.append(acc.astype(BF16))
            ctx = jnp.concatenate(ctx, axis=1)
            o = jnp.dot(ctx, wob[0:NBH * DH, :], preferred_element_type=F32)
            ob[c] = o.astype(BF16)
            ob_send(c, 0).start()
            ob_send(c, 1).start()

    def forward_bulk(c):
        @pl.when(me == 3)
        def _():
            wait_all(ob.at[c], ob_r.at[c])
            ob_send(c, 2).start()

    def wait_q(c):
        @pl.when(me != 1)
        def _():
            wait_all(qb.at[c, pl.ds(0, 4)], q_r.at[c, 0])

        @pl.when(me != 3)
        def _():
            wait_all(qb.at[c, pl.ds(4, 4)], q_r.at[c, 1])

    for c in range(NC):
        wait_q(c)
        if c == 0:
            @pl.when(jnp.logical_not(is_qmaker))
            def _():
                issue_units(2 * NBH, 3 * NBH)

        def bulk_step(h, stat, c=c):
            u = c * NBH + h
            wait_all(kbuf.at[u], ksem.at[u])
            wait_all(vbuf.at[u], vsem.at[u])
            p, inv_l, lse = scores(u, c, h)
            v = vbuf[u].reshape(NG * QB, DH).astype(BF16)
            o = jnp.dot(p, v, preferred_element_type=F32) * inv_l
            po[u] = o.astype(BF16)

            @pl.when(me != 0)
            def _():
                bo_send(c, h).start()

            return jnp.where(sub8 == h, to_row(lse), stat)

        ls[c] = lax.fori_loop(0, NBH, bulk_step, jnp.zeros((8, DH), F32))

        @pl.when(me != 0)
        def _():
            bs_send(c).start()

        if c == 0:
            issue_units(3 * NBH, 4 * NBH)
        elif c == 2:
            issue_units(NBU, NBU + NC)
        elif c == 3:
            issue_units(NBU + NC, NBU + 2 * NC)
        if c >= 1:
            project_bulk(c - 1)
        if c >= 2:
            forward_bulk(c - 2)

    dests = (jnp.where(me == 0, 2, 0), jnp.where(me == 1, 3, 1),
             jnp.where(is_qmaker, 2, 3))
    slots = tuple((d - me + 4) % 4 - 1 for d in dests)

    def ts_send(t, k):
        return remote(lts.at[t], ts.at[t, slots[k]], ts_s.at[t, k],
                      ts_r.at[t], dests[k])

    def to_send(t, k):
        return remote(po.at[NBU + t], to.at[t, slots[k]], to_s.at[t, k],
                      to_r.at[t], dests[k])

    def tail_scores(t, c, h):
        u = NBU + t
        wait_all(kbuf.at[u], ksem.at[u])
        p, inv_l, lse = scores(u, c, h)
        lts[t] = jnp.broadcast_to(to_row(lse), (8, DH))
        for k in range(3):
            ts_send(t, k).start()
        return p, inv_l

    def tail_finish(t, o):
        po[NBU + t] = o.astype(BF16)
        for k in range(3):
            to_send(t, k).start()

    def tail_weights(t):
        wait_all(ts.at[t], ts_r.at[t])
        w = merge_weights([lts[t]] + [ts[t, j] for j in range(3)])
        return [to_col(x[0:1]) for x in w]

    def tail_merge(t, w):
        wait_all(to.at[t], to_r.at[t])
        acc = w[0] * po[NBU + t].astype(F32)
        for j in range(3):
            acc += w[j + 1] * to[t, j].astype(F32)
        return acc.astype(BF16)

    def tail_retire(t):
        ct[t] = tail_merge(t, tail_weights(t))
        for k in range(3):
            ts_send(t, k).wait_send()
            to_send(t, k).wait_send()

    def tail_step(t, carry):
        u = NBU + t
        p, inv_l = tail_scores(t, t % NC, NBH + t // NC)
        wait_all(vbuf.at[u], vsem.at[u])
        v = vbuf[u].reshape(NG * QB, DH).astype(BF16)
        tail_finish(t, jnp.dot(p, v, preferred_element_type=F32) * inv_l)

        @pl.when(t >= TAIL_LAG)
        def _():
            tail_retire(t - TAIL_LAG)

        return carry

    lax.fori_loop(0, 2, tail_step, 0)
    project_bulk(3)
    lax.fori_loop(2, 4, tail_step, 0)
    issue_units(NBU + 2 * NC, NU)
    for i in range(NTH):
        wo_tail_load(i).start()
    forward_bulk(2)
    lax.fori_loop(4, 7, tail_step, 0)
    forward_bulk(3)

    @pl.when(me == 2)
    def _():
        for c in range(NC):
            x_send(c, 0).wait_send()
            x_send(c, 1).wait_send()

    @pl.when(is_qmaker)
    def _():
        for c in range(NC):
            for k in range(3):
                q_send(c, k).wait_send()

    @pl.when(me != 0)
    def _():
        for c in range(NC):
            bs_send(c).wait_send()
            for h in range(NBH):
                bo_send(c, h).wait_send()

    lax.fori_loop(7, NTU - 1, tail_step, 0)

    tl = NTU - 1
    ul = NU - 1
    p, inv_l = tail_scores(tl, NC - 1, NH - 1)
    kp = gp * QB
    o = None
    for i in range(VP):
        piece = vbuf.at[ul, pl.ds(i * gp, gp)]
        wait_all(piece, vpsem.at[i])
        v = piece[...].reshape(kp, DH).astype(BF16)
        oi = jnp.dot(p[:, i * kp:(i + 1) * kp], v, preferred_element_type=F32)
        o = oi if o is None else o + oi
    tail_finish(tl, o * inv_l)

    for t in range(tl - TAIL_LAG, tl):
        tail_retire(t)

    def tail_ctx(i, n):
        return ct[i * NC:i * NC + n].reshape(n * QB, DH)

    def tail_w(i):
        return wof[(NBH + i) * DH:(NBH + i + 1) * DH, :].astype(BF16)

    wo_tail_load(0).wait()
    out_ref[0] = jnp.dot(tail_ctx(0, NC), tail_w(0), preferred_element_type=F32)

    @pl.when(me == 0)
    def _():
        for c in range(NC):
            ob_send(c, 0).wait_send()
            ob_send(c, 1).wait_send()

    @pl.when(me == 3)
    def _():
        for c in range(NC):
            ob_send(c, 2).wait_send()

    @pl.when(jnp.logical_or(me == 1, me == 2))
    def _():
        for c in range(NC):
            wait_all(ob.at[c], ob_r.at[c])

    wo_tail_load(1).wait()
    out_ref[0] += (
        jnp.dot(tail_ctx(1, NC), tail_w(1), preferred_element_type=F32)
        + ob[...].reshape(NC * QB, DM).astype(F32))

    w_last = tail_weights(tl)
    wo_tail_load(2).wait()
    w7 = tail_w(2)
    r3 = (NC - 1) * QB
    out_ref[0, 0:r3, :] += jnp.dot(
        tail_ctx(2, NC - 1), w7, preferred_element_type=F32)
    ctx = tail_merge(tl, w_last)
    out_ref[0, r3:, :] += jnp.dot(ctx, w7, preferred_element_type=F32)
    for k in range(3):
        ts_send(tl, k).wait_send()
        to_send(tl, k).wait_send()


def pallas_dist_sparse_attn_strided_kvseq_b1_sq256_skv4096_hq8_dh128_kernel(
    x: jax.Array,
    Wq: jax.Array,
    K_ext: jax.Array,
    V_ext: jax.Array,
    Wo: jax.Array,
):
    k5 = K_ext.reshape(NG, NC, QB, NH, DH)
    v5 = V_ext.reshape(NG, NC, QB, NH, DH)
    vm = pltpu.VMEM
    dma = pltpu.SemaphoreType.DMA
    scratch = [
        vm((NU, NG, QB, DH), F32),
        vm((NU, NG, QB, DH), F32),
        vm((NC, QB, DM), F32),
        vm((NC, QB, DM), BF16),
        vm((DM, 512), F32),
        vm((DM, 512), BF16),
        vm((DM, DM), F32),
        vm((NBH * DH, DM), BF16),
        vm((NC, NH, QB, DH), BF16),
        vm((NU, QB, DH), BF16),
        vm((NC, 8, DH), F32),
        vm((NC, 3, NBH, QB, DH), BF16),
        vm((NC, 3, 8, DH), F32),
        vm((NTU, 8, DH), F32),
        vm((NTU, 3, QB, DH), BF16),
        vm((NTU, 3, 8, DH), F32),
        vm((NTU, QB, DH), BF16),
        vm((NC, QB, DM), BF16),
        dma((NU,)), dma((NU,)), dma((VP,)),
        dma((NC,)), dma, dma((NTH,)),
        dma((NC, 2)), dma((NC,)),
        dma((NC, 3)), dma((NC, 2)),
        dma((NBU,)), dma((NC,)),
        dma((NC,)), dma((NC,)),
        dma((NC, 3)), dma((NC,)),
        dma((NTU, 3)), dma((NTU,)),
        dma((NTU, 3)), dma((NTU,)),
    ]
    return pl.pallas_call(
        _body,
        out_shape=jax.ShapeDtypeStruct((1, NC * QB, DM), F32),
        in_specs=[pl.BlockSpec(memory_space=pl.ANY)] * 5,
        out_specs=pl.BlockSpec(memory_space=pltpu.VMEM),
        scratch_shapes=scratch,
        compiler_params=pltpu.CompilerParams(
            collective_id=0,
            vmem_limit_bytes=64 * 1024 * 1024,
        ),
    )(x, Wq, k5, v5, Wo)
```

```python
import jax
import jax.numpy as jnp
from jax import lax
from jax.experimental import pallas as pl
from jax.experimental.pallas import tpu as pltpu

NC = 4
QB = 64
NH = 8
DH = 128
DM = 1024
NG = 16
NBH = 5
NTH = NH - NBH
NBU = NC * NBH
NTU = NC * NTH
NU = NBU + NTU
VP = 2
Q_SCALE = 0.08838834764831843 * 1.4426950408889634

F32 = jnp.float32
BF16 = jnp.bfloat16
MESH = pl.DeviceIdType.MESH
NT_DIMS = (((1,), (1,)), ((), ()))

WO_PIECES = ((0, 0, DM), (1, 0, DM // 2), (1, DM // 2, DM),
             (2, 0, DM // 2), (2, DM // 2, DM))

UNITS = [(c, h) for c in range(NC) for h in range(NBH)] + [
    (c, h) for h in range(NBH, NH) for c in range(NC)
]


def _body(
    x_hbm, wq_hbm, k_hbm, v_hbm, wo_hbm, out_ref,
    kbuf, vbuf, xf, xb, wqf, wqb, wof, wob, qb,
    ls, bo, bs, to, ts, ct, ob, wlast,
    ksem, vsem, vpsem, xlsem, wlsem, wtsem,
    xs_s, xs_r, q_s, q_r, bo_s, bo_r, bs_s, bs_r,
    ob_s, ob_r, to_s, to_r, ts_s, ts_r,
):
    me = lax.axis_index("i")
    half = me // 2
    is_qmaker = me % 2 == 1

    def remote(src, dst, ssem, rsem, dev):
        return pltpu.make_async_remote_copy(
            src, dst, ssem, rsem, device_id=(dev,), device_id_type=MESH)

    def wait_all(buf, sem):
        pltpu.make_async_copy(buf, buf, sem).wait()

    gp = NG // VP

    def issue_units(lo, hi):
        for u in range(lo, hi):
            c, h = UNITS[u]
            pltpu.make_async_copy(
                k_hbm.at[:, c, :, h, :], kbuf.at[u], ksem.at[u]).start()
            if u < NU - 1:
                pltpu.make_async_copy(
                    v_hbm.at[:, c, :, h, :], vbuf.at[u], vsem.at[u]).start()
            else:
                for p in range(VP):
                    pltpu.make_async_copy(
                        v_hbm.at[pl.ds(p * gp, gp), c, :, h, :],
                        vbuf.at[u, pl.ds(p * gp, gp)], vpsem.at[p]).start()

    def x_load(c):
        return pltpu.make_async_copy(
            x_hbm.at[0, pl.ds(c * QB, QB), :], xf.at[c], xlsem.at[c])

    def wq_load(hf):
        return pltpu.make_async_copy(
            wq_hbm.at[:, pl.ds(hf * 512, 512)], wqf, wlsem)

    def wo_bulk_load():
        rows = pl.ds(0, NBH * DH)
        return pltpu.make_async_copy(wo_hbm.at[rows], wof.at[rows], wlsem)

    def wo_tail_load(i):
        hd, lo, hi = WO_PIECES[i]
        rows = pl.ds((NBH + hd) * DH, DH)
        cols = pl.ds(lo, hi - lo)
        return pltpu.make_async_copy(
            wo_hbm.at[rows, cols], wof.at[rows, cols], wtsem.at[i])

    @pl.when(me == 2)
    def _():
        for c in range(NC):
            x_load(c).start()

    @pl.when(me == 1)
    def _():
        wq_load(0).start()

    @pl.when(me == 3)
    def _():
        wq_load(1).start()

    @pl.when(me == 0)
    def _():
        wo_bulk_load().start()

    issue_units(0, 2 * NBH)

    barrier = pltpu.get_barrier_semaphore()
    for d in (1, 2, 3):
        pl.semaphore_signal(
            barrier, 1, device_id=((me + d) % 4,), device_id_type=MESH)
    pl.semaphore_wait(barrier, 3)

    def x_send(c, k):
        return remote(xb.at[c], xb.at[c], xs_s.at[c, k], xs_r.at[c], 1 + 2 * k)

    def q_send(c, k):
        rows = qb.at[c, pl.ds(half * 4, 4)]
        dev = (0, 2, 4 - me)[k]
        return remote(rows, rows, q_s.at[c, k], q_r.at[c, half], dev)

    def make_q(c):
        wait_all(xb.at[c], xs_r.at[c])
        q = jnp.dot(xb[c], wqb[...], preferred_element_type=F32) * Q_SCALE
        for i in range(4):
            qb[c, half * 4 + i] = q[:, i * DH:(i + 1) * DH].astype(BF16)
        for k in range(3):
            q_send(c, k).start()

    @pl.when(me == 2)
    def _():
        for c in range(NC):
            x_load(c).wait()
            xb[c] = xf[c].astype(BF16)
            x_send(c, 0).start()
            x_send(c, 1).start()

    @pl.when(is_qmaker)
    def _():
        wq_load(0).wait()
        wqb[...] = wqf[...].astype(BF16)

        def step(c, carry):
            make_q(c)
            return carry

        lax.fori_loop(0, 2, step, 0)

    @pl.when(me == 0)
    def _():
        wo_bulk_load().wait()
        wob[...] = wof[0:NBH * DH, :].astype(BF16)

    row_id = lax.broadcasted_iota(jnp.int32, (QB, DH), 0)
    lane_id = lax.broadcasted_iota(jnp.int32, (QB, DH), 1)
    eye = row_id == lane_id
    eye2 = row_id == lane_id % QB
    sub8 = lax.broadcasted_iota(jnp.int32, (8, DH), 0)

    def to_row(col):
        return jnp.sum(jnp.where(eye2, col, 0.0), axis=0, keepdims=True)

    def to_col(row):
        return jnp.sum(jnp.where(eye, row, 0.0), axis=1, keepdims=True)

    def diag_merge(w, parts):
        lo = lane_id[0:1] < QB
        d = [jnp.where(eye2, jnp.where(lo, w[j], w[j + 1]), 0.0).astype(BF16)
             for j in (0, 2)]
        return jnp.dot(jnp.concatenate(d, axis=1), parts.reshape(4 * QB, DH),
                       preferred_element_type=F32).astype(BF16)

    def scores(u, c, h):
        k = kbuf[u].reshape(NG * QB, DH).astype(BF16)
        s = lax.dot_general(qb[c, h], k, NT_DIMS, preferred_element_type=F32)
        m = jnp.max(s, axis=1, keepdims=True)
        p = jnp.exp2(s - m)
        l = jnp.sum(p, axis=1, keepdims=True)
        return p.astype(BF16), 1.0 / l, m + jnp.log2(l)

    def merge_weights(stats):
        m = jnp.maximum(jnp.maximum(stats[0], stats[1]),
                        jnp.maximum(stats[2], stats[3]))
        e = [jnp.exp2(s - m) for s in stats]
        inv = 1.0 / (e[0] + e[1] + e[2] + e[3])
        return [x * inv for x in e]

    def bo_send(c, h):
        return remote(bo.at[c, h, 3], bo.at[c, h, me - 1], bo_s, bo_r.at[c], 0)

    def bs_send(c):
        return remote(ls.at[c], bs.at[c, me - 1], bs_s, bs_r.at[c], 0)

    def ob_send(c, k):
        return remote(ob.at[c], ob.at[c], ob_s.at[c, k], ob_r.at[c], 1 + 2 * k)

    def ob_fwd(c):
        rows = ob.at[c, half]
        return remote(rows, rows, ob_s.at[c, 0], ob_r.at[c], 2)

    def project_bulk(c):
        wait_all(bs.at[c], bs_r.at[c])
        wait_all(bo.at[c, :, pl.ds(0, 3)], bo_r.at[c])
        w = merge_weights([bs[c, j] for j in range(3)] + [ls[c]])
        ctx = jnp.concatenate(
            [diag_merge([x[h:h + 1] for x in w], bo[c, h]) for h in range(NBH)],
            axis=1)
        o = jnp.dot(ctx, wob[...], preferred_element_type=F32)
        ob[c] = o.astype(BF16).reshape(2, QB // 2, DM)
        ob_send(c, 0).start()
        ob_send(c, 1).start()

    def forward_bulk(c):
        wait_all(ob.at[c], ob_r.at[c])
        ob_fwd(c).start()

    def role_hooks(u):
        pc = (u - (NBH + 1)) // NBH
        fc = (u - 2 * NBH) // NBH

        @pl.when(jnp.logical_and(
            me == 0,
            jnp.logical_and(u == pc * NBH + NBH + 1,
                            jnp.logical_and(u >= NBH + 1, pc < NC))))
        def _():
            project_bulk(pc)

        @pl.when(jnp.logical_and(
            is_qmaker,
            jnp.logical_and(u == fc * NBH + 2 * NBH,
                            jnp.logical_and(u >= 2 * NBH, fc < NC))))
        def _():
            forward_bulk(fc)

    def bulk_step(u, stat):
        c = u // NBH
        h = u % NBH

        @pl.when(jnp.logical_and(h == 0, me != 1))
        def _():
            wait_all(qb.at[c, pl.ds(0, 4)], q_r.at[c, 0])

        @pl.when(jnp.logical_and(h == 0, me != 3))
        def _():
            wait_all(qb.at[c, pl.ds(4, 4)], q_r.at[c, 1])

        @pl.when(u == 0)
        def _():
            issue_units(2 * NBH, 3 * NBH)

        wait_all(kbuf.at[u], ksem.at[u])
        wait_all(vbuf.at[u], vsem.at[u])
        p, inv_l, lse = scores(u, c, h)
        v = vbuf[u].reshape(NG * QB, DH).astype(BF16)
        o = jnp.dot(p, v, preferred_element_type=F32) * inv_l
        bo[c, h, 3] = o.astype(BF16)
        stat = jnp.where(sub8 == h, to_row(lse), stat)
        ls[c] = stat

        @pl.when(me != 0)
        def _():
            bo_send(c, h).start()

        @pl.when(jnp.logical_and(h == NBH - 1, me != 0))
        def _():
            bs_send(c).start()

        @pl.when(u == NBH + 1)
        def _():
            issue_units(3 * NBH, 4 * NBH)

        @pl.when(u == 3 * NBH - 1)
        def _():
            issue_units(NBU, NBU + NC)

        @pl.when(jnp.logical_and(is_qmaker,
                                 jnp.logical_and(h == NBH - 1, c < 2)))
        def _():
            make_q(c + 2)

        role_hooks(u)
        return stat

    lax.fori_loop(0, NBU, bulk_step, jnp.zeros((8, DH), F32))
    issue_units(NBU + NC, NBU + 2 * NC)

    dests = (jnp.where(me == 0, 2, 0), jnp.where(me == 1, 3, 1),
             jnp.where(is_qmaker, 2, 3))
    slots = tuple((d - me + 4) % 4 - 1 for d in dests)

    def ts_send(t, k):
        return remote(ts.at[t, 3], ts.at[t, slots[k]], ts_s, ts_r.at[t],
                      dests[k])

    def to_send(t, k):
        return remote(to.at[t, 3], to.at[t, slots[k]], to_s, to_r.at[t],
                      dests[k])

    def tail_scores(t, c, h):
        u = NBU + t
        wait_all(kbuf.at[u], ksem.at[u])
        p, inv_l, lse = scores(u, c, h)
        ts[t, 3] = to_row(lse)
        for k in range(3):
            ts_send(t, k).start()
        return p, inv_l

    def tail_finish(t, o):
        to[t, 3] = o.astype(BF16)
        for k in range(3):
            to_send(t, k).start()

    def wait_ts(t):
        wait_all(ts.at[t, pl.ds(0, 3)], ts_r.at[t])

    def wait_to(t):
        wait_all(to.at[t, pl.ds(0, 3)], to_r.at[t])

    def tail_weights(t):
        return merge_weights([ts[t, j] for j in range(4)])

    def tail_retire(units):
        for t in units:
            wait_ts(t)
            wait_to(t)
        for t in units:
            ct[t] = diag_merge(tail_weights(t), to[t])

    def tail_step(t, carry):
        u = NBU + t
        p, inv_l = tail_scores(t, t % NC, NBH + t // NC)
        wait_all(vbuf.at[u], vsem.at[u])
        v = vbuf[u].reshape(NG * QB, DH).astype(BF16)
        tail_finish(t, jnp.dot(p, v, preferred_element_type=F32) * inv_l)

        @pl.when(t == NC - 1)
        def _():
            issue_units(NBU + 2 * NC, NU)
            for i in range(len(WO_PIECES)):
                wo_tail_load(i).start()

        role_hooks(u)

        @pl.when(t == 6)
        def _():
            @pl.when(me == 2)
            def _():
                for c in range(NC):
                    x_send(c, 0).wait_send()
                    x_send(c, 1).wait_send()

            @pl.when(is_qmaker)
            def _():
                for c in range(NC):
                    for k in range(3):
                        q_send(c, k).wait_send()

            @pl.when(me != 0)
            def _():
                wait_all(ls, bs_s)
                wait_all(bo.at[:, :, pl.ds(3, 1)], bo_s)

        @pl.when(jnp.logical_or(t == 8, t == 10))
        def _():
            tail_retire([2 * (t - 8) + i for i in range(4)])

        return carry

    lax.fori_loop(0, NTU - 1, tail_step, 0)

    tl = NTU - 1
    ul = NU - 1
    p, inv_l = tail_scores(tl, NC - 1, NH - 1)
    kp = gp * QB
    o = None
    for i in range(VP):
        piece = vbuf.at[ul, pl.ds(i * gp, gp)]
        wait_all(piece, vpsem.at[i])
        v = piece[...].reshape(kp, DH).astype(BF16)
        oi = jnp.dot(p[:, i * kp:(i + 1) * kp], v, preferred_element_type=F32)
        o = oi if o is None else o + oi
    tail_finish(tl, o * inv_l)

    tail_retire([8, 9])

    @pl.when(me == 0)
    def _():
        for c in range(NC):
            ob_send(c, 0).wait_send()
            ob_send(c, 1).wait_send()

    @pl.when(is_qmaker)
    def _():
        for c in range(NC):
            ob_fwd(c).wait_send()

    @pl.when(me == 2)
    def _():
        for c in range(NC):
            wait_all(ob.at[c], ob_r.at[c])

    def tail_ctx(i, n):
        return ct[i * NC:i * NC + n].reshape(n * QB, DH)

    def tail_w(i, lo=0, hi=DM):
        return wof[(NBH + i) * DH:(NBH + i + 1) * DH, lo:hi].astype(BF16)

    wo_tail_load(0).wait()
    out_ref[0] = (
        jnp.dot(tail_ctx(0, NC), tail_w(0), preferred_element_type=F32)
        + ob[...].reshape(NC * QB, DM).astype(F32))

    hc = DM // 2
    r3 = (NC - 1) * QB
    wo_tail_load(1).wait()
    out_ref[0, :, 0:hc] += jnp.dot(
        tail_ctx(1, NC), tail_w(1, 0, hc), preferred_element_type=F32)
    wait_ts(10)
    wait_to(10)
    wo_tail_load(2).wait()
    ct[10] = diag_merge(tail_weights(10), to[10])
    out_ref[0, :, hc:] += jnp.dot(
        tail_ctx(1, NC), tail_w(1, hc, DM), preferred_element_type=F32)

    w_last = None
    for i in range(2):
        if i == 0:
            wait_ts(tl)
        wo_tail_load(3 + i).wait()
        if i == 0:
            w_last = [to_col(x) for x in tail_weights(tl)]
        w7 = tail_w(2, i * hc, (i + 1) * hc)
        wlast[:, i * hc:(i + 1) * hc] = w7
        out_ref[0, 0:r3, i * hc:(i + 1) * hc] += jnp.dot(
            tail_ctx(2, NC - 1), w7, preferred_element_type=F32)
    acc = w_last[3] * to[tl, 3].astype(F32)
    wait_to(tl)
    for j in range(3):
        acc += w_last[j] * to[tl, j].astype(F32)
    out_ref[0, r3:, :] += jnp.dot(
        acc.astype(BF16), wlast[...], preferred_element_type=F32)
    wait_all(ts.at[:, pl.ds(0, 3)], ts_s)
    wait_all(to.at[:, pl.ds(0, 3)], to_s)


def pallas_dist_sparse_attn_strided_kvseq_b1_sq256_skv4096_hq8_dh128_kernel(
    x: jax.Array,
    Wq: jax.Array,
    K_ext: jax.Array,
    V_ext: jax.Array,
    Wo: jax.Array,
):
    k5 = K_ext.reshape(NG, NC, QB, NH, DH)
    v5 = V_ext.reshape(NG, NC, QB, NH, DH)
    vm = pltpu.VMEM
    dma = pltpu.SemaphoreType.DMA
    scratch = [
        vm((NU, NG, QB, DH), F32),
        vm((NU, NG, QB, DH), F32),
        vm((NC, QB, DM), F32),
        vm((NC, QB, DM), BF16),
        vm((DM, 512), F32),
        vm((DM, 512), BF16),
        vm((DM, DM), F32),
        vm((NBH * DH, DM), BF16),
        vm((NC, NH, QB, DH), BF16),
        vm((NC, 8, DH), F32),
        vm((NC, NBH, 4, QB, DH), BF16),
        vm((NC, 3, 8, DH), F32),
        vm((NTU, 4, QB, DH), BF16),
        vm((NTU, 4, 1, DH), F32),
        vm((NTU, QB, DH), BF16),
        vm((NC, 2, QB // 2, DM), BF16),
        vm((DH, DM), BF16),
        dma((NU,)), dma((NU,)), dma((VP,)),
        dma((NC,)), dma, dma((len(WO_PIECES),)),
        dma((NC, 2)), dma((NC,)),
        dma((NC, 3)), dma((NC, 2)),
        dma, dma((NC,)),
        dma, dma((NC,)),
        dma((NC, 2)), dma((NC,)),
        dma, dma((NTU,)),
        dma, dma((NTU,)),
    ]
    return pl.pallas_call(
        _body,
        out_shape=jax.ShapeDtypeStruct((1, NC * QB, DM), F32),
        in_specs=[pl.BlockSpec(memory_space=pl.ANY)] * 5,
        out_specs=pl.BlockSpec(memory_space=pltpu.VMEM),
        scratch_shapes=scratch,
        compiler_params=pltpu.CompilerParams(
            collective_id=0,
            vmem_limit_bytes=64 * 1024 * 1024,
            disable_semaphore_checks=True,
            disable_bounds_checks=True,
        ),
    )(x, Wq, k5, v5, Wo)
```

```python
import jax
import jax.numpy as jnp
from jax import lax
from jax.experimental import pallas as pl
from jax.experimental.pallas import tpu as pltpu

NC = 4
QB = 64
NH = 8
DH = 128
DM = 1024
NG = 16
NBH = 5
NTH = NH - NBH
NBU = NC * NBH
NTU = NC * NTH
NU = NBU + NTU
K_SPLIT = 12
V_SPLIT = 10
Q_SCALE = 0.08838834764831843 * 1.4426950408889634

F32 = jnp.float32
BF16 = jnp.bfloat16
MESH = pl.DeviceIdType.MESH
NT_DIMS = (((1,), (1,)), ((), ()))

WO_PIECES = ((0, 0, 512), (0, 512, DM), (1, 0, 512), (1, 512, DM),
             (2, 0, 512), (2, 512, DM))

MERGE10_AT = 3
ROW_SPLIT = 1
WEIGHTS_AT = 4

UNITS = [(c, h) for c in range(NC) for h in range(NBH)] + [
    (c, h) for h in range(NBH, NH) for c in range(NC)
]


def _body(
    x_hbm, wq_hbm, k_hbm, v_hbm, wo_hbm, out_ref,
    kbuf, vbuf, xf, xb, wqf, wqb, wof, wob, qb,
    ls, bo, bs, to, ts, ct, ob, wlast, pn, oacc, sa, linv, wcol,
    ksem, vsem, vpsem, xlsem, wlsem, wtsem,
    xs_s, xs_r, q_s, q_r, bo_s, bo_r, bs_s, bs_r,
    ob_s, ob_r, to_s, to_r, ts_s, ts_r,
):
    me = lax.axis_index("i")
    half = me // 2
    is_qmaker = me % 2 == 1

    def remote(src, dst, ssem, rsem, dev):
        return pltpu.make_async_remote_copy(
            src, dst, ssem, rsem, device_id=(dev,), device_id_type=MESH)

    def wait_all(buf, sem):
        pltpu.make_async_copy(buf, buf, sem).wait()

    def k_load(u):
        c, h = UNITS[u]
        return pltpu.make_async_copy(
            k_hbm.at[:, c, :, h, :], kbuf.at[u], ksem.at[u])

    def v_load(u):
        c, h = UNITS[u]
        return pltpu.make_async_copy(
            v_hbm.at[:, c, :, h, :], vbuf.at[u], vsem.at[u])

    def last_load(i):
        c, h = UNITS[NU - 1]
        src, dst, cut = ((k_hbm, kbuf, K_SPLIT), (v_hbm, vbuf, V_SPLIT))[i // 2]
        g = pl.ds(cut, NG - cut) if i % 2 else pl.ds(0, cut)
        return pltpu.make_async_copy(
            src.at[g, c, :, h, :], dst.at[NU - 1, g], vpsem.at[i])

    def issue_units(lo, hi):
        for u in range(lo, hi):
            if u < NU - 1:
                k_load(u).start()
                v_load(u).start()
            else:
                for i in range(4):
                    last_load(i).start()

    def x_load(c):
        return pltpu.make_async_copy(
            x_hbm.at[0, pl.ds(c * QB, QB), :], xf.at[c], xlsem.at[c])

    def wq_load(hf):
        return pltpu.make_async_copy(
            wq_hbm.at[:, pl.ds(hf * 512, 512)], wqf, wlsem)

    def wo_bulk_load():
        rows = pl.ds(0, NBH * DH)
        return pltpu.make_async_copy(wo_hbm.at[rows], wof.at[rows], wlsem)

    def wo_tail_load(i):
        hd, lo, hi = WO_PIECES[i]
        rows = pl.ds((NBH + hd) * DH, DH)
        cols = pl.ds(lo, hi - lo)
        return pltpu.make_async_copy(
            wo_hbm.at[rows, cols], wof.at[rows, cols], wtsem.at[i])

    @pl.when(me == 2)
    def _():
        for c in range(NC):
            x_load(c).start()

    @pl.when(me == 1)
    def _():
        wq_load(0).start()

    @pl.when(me == 3)
    def _():
        wq_load(1).start()

    @pl.when(me == 0)
    def _():
        wo_bulk_load().start()

    issue_units(0, 2 * NBH)

    barrier = pltpu.get_barrier_semaphore()
    for d in (1, 2, 3):
        pl.semaphore_signal(
            barrier, 1, device_id=((me + d) % 4,), device_id_type=MESH)
    pl.semaphore_wait(barrier, 3)

    def x_send(c, k):
        return remote(xb.at[c], xb.at[c], xs_s.at[c, k], xs_r.at[c], 1 + 2 * k)

    def q_send(c, k):
        rows = qb.at[c, pl.ds(half * 4, 4)]
        dev = (0, 2, 4 - me)[k]
        return remote(rows, rows, q_s.at[c, k], q_r.at[c, half], dev)

    def make_q(c):
        wait_all(xb.at[c], xs_r.at[c])
        q = jnp.dot(xb[c], wqb[...], preferred_element_type=F32) * Q_SCALE
        for i in range(4):
            qb[c, half * 4 + i] = q[:, i * DH:(i + 1) * DH].astype(BF16)
        for k in range(3):
            q_send(c, k).start()

    @pl.when(me == 2)
    def _():
        for c in range(NC):
            x_load(c).wait()
            xb[c] = xf[c].astype(BF16)
            x_send(c, 0).start()
            x_send(c, 1).start()

    @pl.when(is_qmaker)
    def _():
        wait_all(wqf, wlsem)
        wqb[...] = wqf[...].astype(BF16)

        def step(c, carry):
            make_q(c)
            return carry

        lax.fori_loop(0, 2, step, 0)

    @pl.when(me == 0)
    def _():
        wo_bulk_load().wait()
        wob[...] = wof[0:NBH * DH, :].astype(BF16)

    row_id = lax.broadcasted_iota(jnp.int32, (QB, DH), 0)
    lane_id = lax.broadcasted_iota(jnp.int32, (QB, DH), 1)
    eye = row_id == lane_id
    eye2 = row_id == lane_id % QB
    sub8 = lax.broadcasted_iota(jnp.int32, (8, DH), 0)

    def to_row(col):
        return jnp.sum(jnp.where(eye2, col, 0.0), axis=0, keepdims=True)

    def to_col(row):
        return jnp.sum(jnp.where(eye, row, 0.0), axis=1, keepdims=True)

    def diag_merge(w, parts):
        lo = lane_id[0:1] < QB
        d = [jnp.where(eye2, jnp.where(lo, w[j], w[j + 1]), 0.0).astype(BF16)
             for j in (0, 2)]
        return jnp.dot(jnp.concatenate(d, axis=1), parts.reshape(4 * QB, DH),
                       preferred_element_type=F32).astype(BF16)

    def scores(u, c, h):
        k = kbuf[u].reshape(NG * QB, DH).astype(BF16)
        s = lax.dot_general(qb[c, h], k, NT_DIMS, preferred_element_type=F32)
        m = jnp.max(s, axis=1, keepdims=True)
        p = jnp.exp2(s - m)
        l = jnp.sum(p, axis=1, keepdims=True)
        return p, 1.0 / l, m + jnp.log2(l)

    def merge_weights(stats):
        m = jnp.maximum(jnp.maximum(stats[0], stats[1]),
                        jnp.maximum(stats[2], stats[3]))
        e = [jnp.exp2(s - m) for s in stats]
        inv = 1.0 / (e[0] + e[1] + e[2] + e[3])
        return [x * inv for x in e]

    def bo_send(c, h):
        return remote(bo.at[c, h, 3], bo.at[c, h, me - 1], bo_s, bo_r.at[c], 0)

    def bs_send(c):
        return remote(ls.at[c], bs.at[c, me - 1], bs_s, bs_r.at[c], 0)

    def ob_send(c, k):
        return remote(ob.at[c], ob.at[c], ob_s.at[c, k], ob_r.at[c], 1 + 2 * k)

    def ob_fwd(c):
        rows = ob.at[c, half]
        return remote(rows, rows, ob_s.at[c, 0], ob_r.at[c], 2)

    def project_bulk(c):
        wait_all(bs.at[c], bs_r.at[c])
        wait_all(bo.at[c, :, pl.ds(0, 3)], bo_r.at[c])
        w = merge_weights([bs[c, j] for j in range(3)] + [ls[c]])
        ctx = jnp.concatenate(
            [diag_merge([x[h:h + 1] for x in w], bo[c, h]) for h in range(NBH)],
            axis=1)
        o = jnp.dot(ctx, wob[...], preferred_element_type=F32)
        ob[c] = o.astype(BF16).reshape(2, QB // 2, DM)
        ob_send(c, 0).start()
        ob_send(c, 1).start()

    def forward_bulk(c):
        wait_all(ob.at[c], ob_r.at[c])
        ob_fwd(c).start()

    def role_hooks(u):
        pc = (u - (NBH + 1)) // NBH
        fc = (u - 2 * NBH) // NBH

        @pl.when(jnp.logical_and(
            me == 0,
            jnp.logical_and(u == pc * NBH + NBH + 1,
                            jnp.logical_and(u >= NBH + 1, pc < NC))))
        def _():
            project_bulk(pc)

        @pl.when(jnp.logical_and(
            is_qmaker,
            jnp.logical_and(u == fc * NBH + 2 * NBH,
                            jnp.logical_and(u >= 2 * NBH, fc < NC))))
        def _():
            forward_bulk(fc)

    def bulk_step(u, stat):
        c = u // NBH
        h = u % NBH

        @pl.when(jnp.logical_and(h == 0, me != 1))
        def _():
            wait_all(qb.at[c, pl.ds(0, 4)], q_r.at[c, 0])

        @pl.when(jnp.logical_and(h == 0, me != 3))
        def _():
            wait_all(qb.at[c, pl.ds(4, 4)], q_r.at[c, 1])

        @pl.when(u == 0)
        def _():
            issue_units(2 * NBH, 3 * NBH)

        wait_all(kbuf.at[u], ksem.at[u])
        wait_all(vbuf.at[u], vsem.at[u])
        p, inv_l, lse = scores(u, c, h)
        v = vbuf[u].reshape(NG * QB, DH).astype(BF16)
        o = jnp.dot(p.astype(BF16), v, preferred_element_type=F32) * inv_l
        bo[c, h, 3] = o.astype(BF16)
        stat = jnp.where(sub8 == h, to_row(lse), stat)
        ls[c] = stat

        @pl.when(me != 0)
        def _():
            bo_send(c, h).start()

        @pl.when(jnp.logical_and(h == NBH - 1, me != 0))
        def _():
            bs_send(c).start()

        @pl.when(u == NBH + 1)
        def _():
            issue_units(3 * NBH, 4 * NBH)

        @pl.when(u == 3 * NBH - 1)
        def _():
            issue_units(NBU, NBU + NC)

        @pl.when(jnp.logical_and(is_qmaker,
                                 jnp.logical_and(h == NBH - 1, c < 2)))
        def _():
            make_q(c + 2)

        role_hooks(u)
        return stat

    lax.fori_loop(0, NBU, bulk_step, jnp.zeros((8, DH), F32))
    issue_units(NBU + NC, NBU + 2 * NC)

    dests = (jnp.where(me == 0, 2, 0), jnp.where(me == 1, 3, 1),
             jnp.where(is_qmaker, 2, 3))
    slots = tuple((d - me + 4) % 4 - 1 for d in dests)

    def ts_send(t, k):
        return remote(ts.at[t, 3], ts.at[t, slots[k]], ts_s, ts_r.at[t],
                      dests[k])

    def to_send(t, k):
        return remote(to.at[t, 3], to.at[t, slots[k]], to_s, to_r.at[t],
                      dests[k])

    def tail_scores(t, c, h):
        u = NBU + t
        wait_all(kbuf.at[u], ksem.at[u])
        p, inv_l, lse = scores(u, c, h)
        ts[t, 3] = to_row(lse)
        for k in range(3):
            ts_send(t, k).start()
        return p.astype(BF16), inv_l

    def tail_finish(t, o):
        to[t, 3] = o.astype(BF16)
        for k in range(3):
            to_send(t, k).start()

    def wait_ts(t):
        wait_all(ts.at[t, pl.ds(0, 3)], ts_r.at[t])

    def wait_to(t):
        wait_all(to.at[t, pl.ds(0, 3)], to_r.at[t])

    def tail_weights(t):
        return merge_weights([ts[t, j] for j in range(4)])

    def tail_retire(units):
        for t in units:
            wait_ts(t)
            wait_to(t)
        for t in units:
            ct[t] = diag_merge(tail_weights(t), to[t])

    def tail_step(t, carry):
        u = NBU + t
        p, inv_l = tail_scores(t, t % NC, NBH + t // NC)
        wait_all(vbuf.at[u], vsem.at[u])
        v = vbuf[u].reshape(NG * QB, DH).astype(BF16)
        tail_finish(t, jnp.dot(p, v, preferred_element_type=F32) * inv_l)

        @pl.when(t == NC - 1)
        def _():
            issue_units(NBU + 2 * NC, NU)
            for i in range(len(WO_PIECES)):
                wo_tail_load(i).start()

        role_hooks(u)

        @pl.when(t == 6)
        def _():
            @pl.when(me == 2)
            def _():
                for c in range(NC):
                    x_send(c, 0).wait_send()
                    x_send(c, 1).wait_send()

            @pl.when(is_qmaker)
            def _():
                for c in range(NC):
                    for k in range(3):
                        q_send(c, k).wait_send()

            @pl.when(me != 0)
            def _():
                wait_all(ls, bs_s)
                wait_all(bo.at[:, :, pl.ds(3, 1)], bo_s)

        @pl.when(jnp.logical_or(t == 7, t == 9))
        def _():
            tail_retire([(t - 7) * 3 // 2 + i for i in range(3)])

        return carry

    tl = NTU - 1
    ul = NU - 1
    lax.fori_loop(0, tl, tail_step, 0)

    def blocks(buf, lo, hi):
        return buf[ul, lo:hi].reshape((hi - lo) * QB, DH).astype(BF16)

    q = qb[NC - 1, NH - 1]
    last_load(0).wait()
    sa[...] = lax.dot_general(q, blocks(kbuf, 0, K_SPLIT), NT_DIMS,
                              preferred_element_type=F32)
    last_load(1).wait()
    s = jnp.concatenate(
        [sa[...], lax.dot_general(q, blocks(kbuf, K_SPLIT, NG), NT_DIMS,
                                  preferred_element_type=F32)], axis=1)
    m = jnp.max(s, axis=1, keepdims=True)
    p = jnp.exp2(s - m)
    pn[...] = p.astype(BF16)
    l = jnp.sum(p, axis=1, keepdims=True)
    last_load(2).wait()
    oacc[...] = jnp.dot(pn[:, 0:V_SPLIT * QB], blocks(vbuf, 0, V_SPLIT),
                        preferred_element_type=F32)
    linv[...] = jnp.broadcast_to(1.0 / l, (QB, DH))
    ts[tl, 3] = to_row(m + jnp.log2(l))
    for k in range(3):
        ts_send(tl, k).start()
    last_load(3).wait()
    o = oacc[...] + jnp.dot(pn[:, V_SPLIT * QB:], blocks(vbuf, V_SPLIT, NG),
                            preferred_element_type=F32)
    tail_finish(tl, o * linv[...])

    tail_retire([6, 7, 8, 9])

    @pl.when(me == 0)
    def _():
        for c in range(NC):
            ob_send(c, 0).wait_send()
            ob_send(c, 1).wait_send()

    @pl.when(is_qmaker)
    def _():
        for c in range(NC):
            ob_fwd(c).wait_send()

    @pl.when(me == 2)
    def _():
        for c in range(NC):
            wait_all(ob.at[c], ob_r.at[c])

    def tail_ctx(i, n):
        return ct[i * NC:i * NC + n].reshape(n * QB, DH)

    def tail_w(i, lo=0, hi=DM):
        return wof[(NBH + i) * DH:(NBH + i + 1) * DH, lo:hi].astype(BF16)

    r3 = (NC - 1) * QB
    w_last = None
    n_wo = len(WO_PIECES)
    for i, (hd, lo, hi) in enumerate(WO_PIECES):
        if i == MERGE10_AT:
            wait_ts(10)
            wait_to(10)
        if i == WEIGHTS_AT:
            wait_ts(tl)
        wo_tail_load(i).wait()
        if i == MERGE10_AT:
            ct[10] = diag_merge(tail_weights(10), to[10])
        if i == WEIGHTS_AT:
            for j, x in enumerate(tail_weights(tl)):
                wcol[j] = jnp.broadcast_to(to_col(x), (QB, DH))
        w = tail_w(hd, lo, hi)
        if hd == 0:
            out_ref[0, :, lo:hi] = (
                jnp.dot(tail_ctx(0, NC), w, preferred_element_type=F32)
                + ob[:, :, :, lo:hi].reshape(NC * QB, hi - lo).astype(F32))
        elif hd < NTH - 1:
            out_ref[0, :, lo:hi] += jnp.dot(
                tail_ctx(hd, NC), w, preferred_element_type=F32)
        else:
            wlast[:, lo:hi] = w
            cx = tail_ctx(hd, NC - 1)
            rs = r3 // ROW_SPLIT
            for r in range(ROW_SPLIT):
                out_ref[0, r * rs:(r + 1) * rs, lo:hi] += jnp.dot(
                    cx[r * rs:(r + 1) * rs], w, preferred_element_type=F32)
    wait_to(tl)
    acc = wcol[0] * to[tl, 0].astype(F32)
    for j in range(1, 4):
        acc += wcol[j] * to[tl, j].astype(F32)
    out_ref[0, r3:, :] += jnp.dot(
        acc.astype(BF16), wlast[...], preferred_element_type=F32)
    wait_all(ts.at[:, pl.ds(0, 3)], ts_s)
    wait_all(to.at[:, pl.ds(0, 3)], to_s)


def pallas_dist_sparse_attn_strided_kvseq_b1_sq256_skv4096_hq8_dh128_kernel(
    x: jax.Array,
    Wq: jax.Array,
    K_ext: jax.Array,
    V_ext: jax.Array,
    Wo: jax.Array,
):
    k5 = K_ext.reshape(NG, NC, QB, NH, DH)
    v5 = V_ext.reshape(NG, NC, QB, NH, DH)
    vm = pltpu.VMEM
    dma = pltpu.SemaphoreType.DMA
    scratch = [
        vm((NU, NG, QB, DH), F32),
        vm((NU, NG, QB, DH), F32),
        vm((NC, QB, DM), F32),
        vm((NC, QB, DM), BF16),
        vm((DM, 512), F32),
        vm((DM, 512), BF16),
        vm((DM, DM), F32),
        vm((NBH * DH, DM), BF16),
        vm((NC, NH, QB, DH), BF16),
        vm((NC, 8, DH), F32),
        vm((NC, NBH, 4, QB, DH), BF16),
        vm((NC, 3, 8, DH), F32),
        vm((NTU, 4, QB, DH), BF16),
        vm((NTU, 4, 1, DH), F32),
        vm((NTU, QB, DH), BF16),
        vm((NC, 2, QB // 2, DM), BF16),
        vm((DH, DM), BF16),
        vm((QB, NG * QB), BF16),
        vm((QB, DH), F32),
        vm((QB, K_SPLIT * QB), F32),
        vm((QB, DH), F32),
        vm((4, QB, DH), F32),
        dma((NU,)), dma((NU,)), dma((4,)),
        dma((NC,)), dma, dma((len(WO_PIECES),)),
        dma((NC, 2)), dma((NC,)),
        dma((NC, 3)), dma((NC, 2)),
        dma, dma((NC,)),
        dma, dma((NC,)),
        dma((NC, 2)), dma((NC,)),
        dma, dma((NTU,)),
        dma, dma((NTU,)),
    ]
    return pl.pallas_call(
        _body,
        out_shape=jax.ShapeDtypeStruct((1, NC * QB, DM), F32),
        in_specs=[pl.BlockSpec(memory_space=pl.ANY)] * 5,
        out_specs=pl.BlockSpec(memory_space=pltpu.VMEM),
        scratch_shapes=scratch,
        compiler_params=pltpu.CompilerParams(
            collective_id=0,
            vmem_limit_bytes=64 * 1024 * 1024,
            disable_semaphore_checks=False,
            disable_bounds_checks=False,
        ),
    )(x, Wq, k5, v5, Wo)
```

```python
import functools

import jax
import jax.numpy as jnp
from jax import lax
from jax.experimental import pallas as pl
from jax.experimental.pallas import tpu as pltpu

NC = 4
QB = 64
NH = 8
DH = 128
DM = 1024
NG = 16
NBH = 5
NTH = NH - NBH
NBU = NC * NBH
NTU = NC * NTH
NU = NBU + NTU
Q_SCALE = 0.08838834764831843 * 1.4426950408889634

F32 = jnp.float32
BF16 = jnp.bfloat16
MESH = pl.DeviceIdType.MESH
NT_DIMS = (((1,), (1,)), ((), ()))

UNITS = [(c, h) for c in range(NC) for h in range(NBH)] + [
    (c, h) for h in range(NBH, NH) for c in range(NC)
]

PARTS = 2
AHEAD = 5
K_SPLIT = 12
V_SPLIT = 10
N_FLY = 7
FLY_LAG = 3
WO_STEP = 29
WO_PIECES = ((0, 0, 512), (0, 512, DM), (1, 0, 512), (1, 512, DM),
             (2, 0, 512), (2, 512, DM))
MERGE_AT = ((4, 5), (6, 7), (8, 9), (10,), (), ())
WEIGHTS_AT = 4

N_PRE = 5
STEP0 = 2 + N_PRE
N_SLOT = STEP0 + NU
X_SLOTS = {2: 2, 3: 4}
MAKEQ_SLOTS = (2, 4, 6, 10)
RELAY_SLOTS = (5, 9, 13, 18)
PROJECT_STEPS = (12, 15, 18, 21)
SECOND_STEPS = (13, 16, 19, 23)
FORWARD_STEPS = (16, 19, 22, 25)
ACT_X, ACT_MAKEQ, ACT_RELAY, ACT_PROJECT, ACT_SECOND, ACT_FORWARD = range(6)

SWAPS = "SSSS-+S-S+BS+S-S+BS+S-S+-S+S"
PERMS = {"+": (1, 2, 3, 0), "-": (3, 0, 1, 2), "B": (3, 2, 1, 0)}
MARKS = {".": "..", "u": "u.", "d": "d.", "U": "uu", "D": "dd", "b": "ud"}
PLANS = (
    "ud.dudu" ".d.u..dudududu.dudud" "duud.duu....",
    "ddu.ddu" "d.u..u.uduuuuu.uuudu" "dudu.duu....",
    "......." "..DU.D.UDuudduudbud." "dudu.duu....",
    "uud.udu" "d.d..u.uduuduuuu.uud" "duudd.uu....",
)
MARGIN = 3
STAGE_FIRST = 3
STAGE_IN = (
    "0121101" "01100101011011110111" "011101110000",
    "1012110" "10101010100111011110" "111011110000",
    "0101210" "00101010111101111101" "111011110000",
    "1012110" "01110001101011011110" "111011110000",
)
STAGE_OUT = (
    "2101120" "10010101011110111101" "110111011100",
    "0310111" "11010101001101110111" "101110111100",
    "0031011" "01010101011111011111" "011110111100",
    "0310111" "20001110001110110111" "101110111100",
)
STAGE_MARGIN = 1
RING = 16


def _push_table(chip):
    first = NU - len(SWAPS)
    todo = {"u": [], "d": []}
    for i, name in enumerate(SWAPS):
        if name == "S":
            continue
        dest = PERMS[name][chip]
        way = "u" if dest == (chip + 1) % 4 else "d"
        c, h = UNITS[first + i]
        for is_v in range(2):
            code = ((((first + i) * NC + c) * NH + h) * 2 + is_v) * 4 + dest
            todo[way].append((first + i, code))
    table = []
    assert len(PLANS[chip]) == N_SLOT
    for slot, mark in enumerate(PLANS[chip]):
        for way in MARKS[mark]:
            if way == ".":
                table.append(-1)
            else:
                u, code = todo[way].pop(0)
                assert slot - STEP0 <= u - MARGIN, (chip, slot, u)
                table.append(code)
    assert not todo["u"] and not todo["d"], (chip, todo)
    return table


def _staged_units():
    first = NU - len(SWAPS)
    return [first + i for i, name in enumerate(SWAPS) if name == "S"]


def _wait_slot(u):
    return 2 + u if u < N_PRE else STEP0 + u


def _stage_table(chip):
    units = _staged_units()
    n_in, n_out = STAGE_FIRST, 0
    table = []
    for slot in range(N_SLOT):
        a, b = int(STAGE_IN[chip][slot]), int(STAGE_OUT[chip][slot])
        assert n_out + b <= n_in, (chip, slot)
        for j in range(n_out, n_out + b):
            due = _wait_slot(units[j // 2])
            assert slot <= due - STAGE_MARGIN, (chip, slot, j)
        for j in range(max(n_in, RING), n_in + a):
            assert slot >= _wait_slot(units[(j - RING) // 2]), (chip, slot, j)
        table.append(n_in | (n_in + a) << 6 | n_out << 12 | (n_out + b) << 18)
        n_in += a
        n_out += b
    assert n_in == n_out == 2 * len(units), (chip, n_in, n_out)
    return table


def _action_table(chip):
    def steps(when):
        return [(STEP0 + st, c) for c, st in enumerate(when)]

    events = {}
    if chip == 0:
        events[ACT_RELAY] = list(zip(RELAY_SLOTS, range(NC)))
        events[ACT_PROJECT] = steps(PROJECT_STEPS)
        events[ACT_SECOND] = steps(SECOND_STEPS)
    elif chip == 2:
        events[ACT_X] = [(slot, c) for c, slot in X_SLOTS.items()]
    else:
        events[ACT_MAKEQ] = list(zip(MAKEQ_SLOTS, range(NC)))
        events[ACT_FORWARD] = steps(FORWARD_STEPS)
    table = [0] * N_SLOT
    for act, items in events.items():
        for slot, c in items:
            table[slot] |= (c + 1) << (3 * act)
    return table


def _body(
    x_hbm, wq_hbm, k_hbm, v_hbm, wo_hbm, out_ref,
    kbuf, vbuf, xf, xb, wqf, wqb, wof, wob, qb,
    ls, bo, bs, to, ts, ct, ob, wlast, pn, oacc, sa, linv, wcol,
    ptab, atab, utab, gtab, stab, stage,
    ksem, vsem, lsem, xlsem, wlsem, wtsem,
    xs_s, xs_r, q_s, q_r, bo_s, bo_r, bs_s, bs_r,
    ob_s, ob_r, to_s, to_r, ts_s, ts_r, sw_s, fo_r, fs_r, st_s,
):
    me = lax.axis_index("i")
    half = me // 2
    is_qmaker = me % 2 == 1
    staged = _staged_units()
    n_swap = len(SWAPS) - len(staged)
    first = NU - len(SWAPS)
    kv = ((k_hbm, kbuf, ksem), (v_hbm, vbuf, vsem))

    def remote(src, dst, ssem, rsem, dev):
        return pltpu.make_async_remote_copy(
            src, dst, ssem, rsem, device_id=(dev,), device_id_type=MESH)

    def wait_all(buf, sem):
        pltpu.make_async_copy(buf, buf, sem).wait()

    def load_blocks(u, c, h, is_v, lo, hi, sem):
        src, dst, _ = kv[is_v]
        g = pl.ds(lo, hi - lo)
        for r in range(PARTS):
            keys = pl.ds(r * (QB // PARTS), QB // PARTS)
            pltpu.make_async_copy(
                src.at[g, c, keys, h, :], dst.at[u, g, keys], sem).start()

    def load_unit(u, c, h, lo):
        for is_v in range(2):
            load_blocks(u, c, h, is_v, lo, NG, kv[is_v][2].at[u])

    def unit_of(u):
        word = utab[u]
        return word >> 3, word & 7

    def load_ahead(u):
        load_unit(u, *unit_of(u), 1)

    def load_last():
        u = NU - 1
        c, h = UNITS[u]
        for is_v, cut in enumerate((K_SPLIT, V_SPLIT)):
            load_blocks(u, c, h, is_v, 1, cut, kv[is_v][2].at[u])
            load_blocks(u, c, h, is_v, cut, NG, lsem.at[is_v])

    def last_wait(is_v, piece):
        cut = (K_SPLIT, V_SPLIT)[is_v]
        _, buf, sem = kv[is_v]
        if piece == 0:
            wait_all(buf.at[NU - 1, pl.ds(0, cut)], sem.at[NU - 1])
        else:
            wait_all(buf.at[NU - 1, pl.ds(cut, NG - cut)], lsem.at[is_v])

    def wait_unit(u):
        wait_all(kbuf.at[u], ksem.at[u])
        wait_all(vbuf.at[u], vsem.at[u])

    def push(slot, which=(0, 1)):
        for i in which:
            code = ptab[2 * slot + i]
            for is_v in range(2):
                @pl.when(jnp.logical_and(code >= 0, ((code >> 2) & 1) == is_v))
                def _(is_v=is_v, code=code):
                    src, dst, sem = kv[is_v]
                    u = code >> 8
                    block = src.at[0, (code >> 6) & 3, :, (code >> 3) & 7, :]
                    remote(block, dst.at[u, 0], sw_s, sem.at[u],
                           code & 3).start()

    def stage_in(j, c, h, is_v):
        pltpu.make_async_copy(
            kv[is_v][0].at[0, c, :, h, :], stage.at[j & (RING - 1)],
            st_s.at[j]).start()

    def stage_step(slot):
        word = gtab[slot]

        def drain(j, carry):
            u = stab[j >> 1]
            block = stage.at[j & (RING - 1)]
            wait_all(block, st_s.at[j])
            for is_v in range(2):
                @pl.when((j & 1) == is_v)
                def _(is_v=is_v):
                    _, dst, sem = kv[is_v]
                    pltpu.make_async_copy(
                        block, dst.at[u, 0], sem.at[u]).start()
            return carry

        def fetch(j, carry):
            c, h = unit_of(stab[j >> 1])
            for is_v in range(2):
                @pl.when((j & 1) == is_v)
                def _(is_v=is_v):
                    stage_in(j, c, h, is_v)
            return carry

        lax.fori_loop((word >> 12) & 63, (word >> 18) & 63, drain, 0)
        lax.fori_loop(word & 63, (word >> 6) & 63, fetch, 0)

    def action(slot, act, fn):
        field = (atab[slot] >> (3 * act)) & 7

        @pl.when(field > 0)
        def _():
            fn(field - 1)

    def x_load(c):
        return pltpu.make_async_copy(
            x_hbm.at[0, pl.ds(c * QB, QB), :], xf.at[c], xlsem.at[c])

    def wq_load(hf):
        return pltpu.make_async_copy(
            wq_hbm.at[:, pl.ds(hf * 512, 512)], wqf, wlsem)

    def wo_bulk_load():
        rows = pl.ds(0, NBH * DH)
        return pltpu.make_async_copy(wo_hbm.at[rows], wof.at[rows], wlsem)

    def wo_tail_load(i):
        hd, lo, hi = WO_PIECES[i]
        rows = pl.ds((NBH + hd) * DH, DH)
        cols = pl.ds(lo, hi - lo)
        return pltpu.make_async_copy(
            wo_hbm.at[rows, cols], wof.at[rows, cols], wtsem.at[i])

    def send_x(c):
        for k in range(2):
            remote(xb.at[c], xb.at[c], xs_s.at[k], xs_r.at[c],
                   1 + 2 * k).start()

    def wait_q(c, k):
        wait_all(qb.at[c, pl.ds(k * 4, 4)], q_r.at[c, k])

    def make_q(c):
        wait_all(xb.at[c], xs_r.at[c])
        q = jnp.dot(xb[c], wqb[...], preferred_element_type=F32) * Q_SCALE
        for i in range(4):
            qb[c, half * 4 + i] = q[:, i * DH:(i + 1) * DH].astype(BF16)
        rows = qb.at[c, pl.ds(half * 4, 4)]
        for k in range(2):
            remote(rows, rows, q_s.at[k], q_r.at[c, half], 2 * k).start()

    def relay_q(c):
        for k in range(2):
            wait_q(c, k)
            rows = qb.at[c, pl.ds(k * 4, 4)]
            remote(rows, rows, q_s.at[k], q_r.at[c, k], 3 - 2 * k).start()

    def q_hooks(slot):
        action(slot, ACT_MAKEQ, make_q)
        action(slot, ACT_RELAY, relay_q)

    @pl.when(me == 2)
    def _():
        for c in range(NC):
            x_load(c).start()

    @pl.when(me == 1)
    def _():
        wq_load(0).start()

    @pl.when(me == 3)
    def _():
        wq_load(1).start()

    @pl.when(me == 0)
    def _():
        wo_bulk_load().start()

    for j in range(STAGE_FIRST):
        stage_in(j, *UNITS[staged[j // 2]], j % 2)

    assert first <= AHEAD
    for u in range(AHEAD):
        load_unit(u, *UNITS[u], int(u >= first))

    barrier = pltpu.get_barrier_semaphore()
    for d in (1, 2, 3):
        pl.semaphore_signal(
            barrier, 1, device_id=((me + d) % 4,), device_id_type=MESH)

    def fill(ref, tables):
        for i, words in enumerate(zip(*tables)):
            word = jnp.int32(words[0])
            for chip in range(1, 4):
                if words[chip] != words[0]:
                    word = jnp.where(me == chip, words[chip], word)
            ref[i] = word

    fill(ptab, [_push_table(chip) for chip in range(4)])
    fill(atab, [_action_table(chip) for chip in range(4)])
    fill(gtab, [_stage_table(chip) for chip in range(4)])
    fill(utab, [[c * NH + h for c, h in UNITS]] * 4)
    fill(stab, [staged] * 4)

    pl.semaphore_wait(barrier, 3)

    @pl.when(me == 2)
    def _():
        x_load(0).wait()
        xb[0] = xf[0].astype(BF16)
        send_x(0)

    push(0)
    stage_step(0)

    @pl.when(is_qmaker)
    def _():
        wait_all(wqf, wlsem)

    @pl.when(me == 0)
    def _():
        wo_bulk_load().wait()

    push(1)
    stage_step(1)

    @pl.when(me == 2)
    def _():
        for c in range(1, NC):
            x_load(c).wait()
            xb[c] = xf[c].astype(BF16)
        send_x(1)

    @pl.when(is_qmaker)
    def _():
        wqb[...] = wqf[...].astype(BF16)

    @pl.when(me == 0)
    def _():
        wob[...] = wof[0:NBH * DH, :].astype(BF16)

    def pre_step(u, carry):
        wait_unit(u)
        load_ahead(u + AHEAD)
        push(2 + u)
        stage_step(2 + u)
        action(2 + u, ACT_X, send_x)
        q_hooks(2 + u)
        return carry

    lax.fori_loop(0, N_PRE, pre_step, 0)

    row_id = lax.broadcasted_iota(jnp.int32, (QB, DH), 0)
    lane_id = lax.broadcasted_iota(jnp.int32, (QB, DH), 1)
    eye = row_id == lane_id
    eye2 = row_id == lane_id % QB
    sub8 = lax.broadcasted_iota(jnp.int32, (8, DH), 0)

    def to_row(col):
        return jnp.sum(jnp.where(eye2, col, 0.0), axis=0, keepdims=True)

    def to_col(row):
        return jnp.sum(jnp.where(eye, row, 0.0), axis=1, keepdims=True)

    def scores(u, c, h):
        k = kbuf[u].reshape(NG * QB, DH).astype(BF16)
        s = lax.dot_general(qb[c, h], k, NT_DIMS, preferred_element_type=F32)
        m = jnp.max(s, axis=1, keepdims=True)
        p = jnp.exp2(s - m)
        l = jnp.sum(p, axis=1, keepdims=True)
        return p.astype(BF16), 1.0 / l, m + jnp.log2(l)

    def merge_weights(stats):
        m = functools.reduce(jnp.maximum, stats)
        e = [jnp.exp2(s - m) for s in stats]
        total = functools.reduce(jnp.add, e)
        inv = 1.0 / total
        return [x * inv for x in e], m + jnp.log2(total)

    def diag_merge(w, parts):
        lo = lane_id[0:1] < QB
        d = [jnp.where(eye2, jnp.where(lo, w[j], w[j + 1]), 0.0).astype(BF16)
             for j in range(0, len(w), 2)]
        return jnp.dot(jnp.concatenate(d, axis=1),
                       parts.reshape(len(w) * QB, DH),
                       preferred_element_type=F32).astype(BF16)

    def ob_send(c, rnd):
        for k in range(2):
            hf = k ^ rnd
            rows = ob.at[c, hf]
            remote(rows, rows, ob_s.at[k], ob_r.at[c, hf], 1 + 2 * k).start()

    def ob_wait(c, hf):
        wait_all(ob.at[c, hf], ob_r.at[c, hf])

    def project_bulk(c):
        wait_all(bs.at[c], bs_r.at[c])
        wait_all(bo.at[c, :, pl.ds(0, 3)], bo_r.at[c])
        w, _ = merge_weights([bs[c, j] for j in range(3)] + [ls[c]])
        ctx = jnp.concatenate(
            [diag_merge([x[h:h + 1] for x in w], bo[c, h]) for h in range(NBH)],
            axis=1)
        o = jnp.dot(ctx, wob[...], preferred_element_type=F32)
        ob[c] = o.astype(BF16).reshape(2, QB // 2, DM)
        ob_send(c, 0)

    def forward_bulk(c):
        ob_wait(c, half)
        rows = ob.at[c, half]
        remote(rows, rows, ob_s.at[0], ob_r.at[c, half], 2).start()

    def role_hooks(slot):
        action(slot, ACT_PROJECT, project_bulk)
        action(slot, ACT_SECOND, lambda c: ob_send(c, 1))
        action(slot, ACT_FORWARD, forward_bulk)

    def bulk_step(u, stat):
        slot = STEP0 + u
        c, h = unit_of(u)

        @pl.when(jnp.logical_and(h == 0, me >= 2))
        def _():
            wait_q(c, 0)

        @pl.when(jnp.logical_and(h == 0, jnp.logical_or(me == 1, me == 2)))
        def _():
            wait_q(c, 1)

        @pl.when(u >= N_PRE)
        def _():
            wait_unit(u)
            load_ahead(u + AHEAD)

        push(slot, (0,))
        p, inv_l, lse = scores(u, c, h)
        v = vbuf[u].reshape(NG * QB, DH).astype(BF16)
        o = jnp.dot(p, v, preferred_element_type=F32) * inv_l
        bo[c, h, 3] = o.astype(BF16)
        stat = jnp.where(sub8 == h, to_row(lse), stat)
        ls[c] = stat

        @pl.when(me != 0)
        def _():
            remote(bo.at[c, h, 3], bo.at[c, h, me - 1], bo_s, bo_r.at[c],
                   0).start()

        @pl.when(jnp.logical_and(h == NBH - 1, me != 0))
        def _():
            remote(ls.at[c], bs.at[c, me - 1], bs_s, bs_r.at[c], 0).start()

        push(slot, (1,))
        stage_step(slot)
        q_hooks(slot)
        role_hooks(slot)
        return stat

    lax.fori_loop(0, NBU, bulk_step, jnp.zeros((8, DH), F32))

    dests = (jnp.where(me == 0, 2, 0), jnp.where(me == 1, 3, 1),
             jnp.where(is_qmaker, 2, 3))
    slots = tuple((d - me + 4) % 4 - 1 for d in dests)

    def gather_send(buf, t, ssem, rsem):
        for k in range(3):
            remote(buf.at[t, 3], buf.at[t, slots[k]], ssem.at[1], rsem.at[t],
                   dests[k]).start()

    def wait_ts(t):
        wait_all(ts.at[t, pl.ds(0, 3)], ts_r.at[t])

    def wait_to(t):
        wait_all(to.at[t, pl.ds(0, 3)], to_r.at[t])

    def tail_weights(t):
        return merge_weights([ts[t, j] for j in range(4)])[0]

    def fly_send(t, rnd):
        dev = jnp.where(((t + rnd) & 1) == 0, me ^ 1, 3 - me)
        src = 3 - 2 * rnd
        remote(ts.at[t, src], ts.at[t, src - 1], ts_s.at[0], fs_r.at[t, rnd],
               dev).start()
        remote(to.at[t, src], to.at[t, src - 1], to_s.at[0], fo_r.at[t, rnd],
               dev).start()

    def fly_wait(t, rnd):
        dst = 2 - 2 * rnd
        wait_all(ts.at[t, dst], fs_r.at[t, rnd])
        wait_all(to.at[t, dst], fo_r.at[t, rnd])

    def fly_merge(t, rnd):
        lo = 2 - 2 * rnd
        w, lse = merge_weights([ts[t, lo], ts[t, lo + 1]])
        return diag_merge(w, to[t, lo:lo + 2]), lse

    def tail_step(t, carry):
        u = NBU + t
        slot = STEP0 + u
        wait_all(kbuf.at[u], ksem.at[u])
        p, inv_l, lse = scores(u, *unit_of(u))
        ts[t, 3] = to_row(lse)

        @pl.when(t >= N_FLY)
        def _():
            gather_send(ts, t, ts_s, ts_r)

        push(slot, (0,))
        wait_all(vbuf.at[u], vsem.at[u])
        v = vbuf[u].reshape(NG * QB, DH).astype(BF16)
        o = jnp.dot(p, v, preferred_element_type=F32) * inv_l
        to[t, 3] = o.astype(BF16)

        @pl.when(t >= N_FLY)
        def _():
            gather_send(to, t, to_s, to_r)

        @pl.when(t < N_FLY)
        def _():
            fly_send(t, 0)

        @pl.when(jnp.logical_and(t >= FLY_LAG, t < N_FLY + FLY_LAG))
        def _():
            f = t - FLY_LAG
            fly_wait(f, 0)
            to[f, 1], ts[f, 1] = fly_merge(f, 0)
            fly_send(f, 1)

        push(slot, (1,))
        stage_step(slot)

        @pl.when(u + AHEAD < NU - 1)
        def _():
            load_ahead(u + AHEAD)

        @pl.when(u + AHEAD == NU - 1)
        def _():
            load_last()

        @pl.when(u == WO_STEP)
        def _():
            for i in range(len(WO_PIECES)):
                wo_tail_load(i).start()

        role_hooks(slot)

        @pl.when(jnp.logical_and(t >= 2 * FLY_LAG,
                                 t - 2 * FLY_LAG < MERGE_AT[0][0]))
        def _():
            f = t - 2 * FLY_LAG
            fly_wait(f, 1)
            ct[f] = fly_merge(f, 1)[0]

        return carry

    tl = NTU - 1
    lax.fori_loop(0, tl, tail_step, 0)

    def blocks(buf, lo, hi):
        return buf[NU - 1, lo:hi].reshape((hi - lo) * QB, DH).astype(BF16)

    q = qb[NC - 1, NH - 1]
    last_wait(0, 0)
    sa[...] = lax.dot_general(q, blocks(kbuf, 0, K_SPLIT), NT_DIMS,
                              preferred_element_type=F32)
    last_wait(0, 1)
    s = jnp.concatenate(
        [sa[...], lax.dot_general(q, blocks(kbuf, K_SPLIT, NG), NT_DIMS,
                                  preferred_element_type=F32)], axis=1)
    m = jnp.max(s, axis=1, keepdims=True)
    p = jnp.exp2(s - m)
    pn[...] = p.astype(BF16)
    l = jnp.sum(p, axis=1, keepdims=True)
    last_wait(1, 0)
    oacc[...] = jnp.dot(pn[:, 0:V_SPLIT * QB], blocks(vbuf, 0, V_SPLIT),
                        preferred_element_type=F32)
    linv[...] = jnp.broadcast_to(1.0 / l, (QB, DH))
    ts[tl, 3] = to_row(m + jnp.log2(l))
    gather_send(ts, tl, ts_s, ts_r)
    last_wait(1, 1)
    o = oacc[...] + jnp.dot(pn[:, V_SPLIT * QB:], blocks(vbuf, V_SPLIT, NG),
                            preferred_element_type=F32)
    to[tl, 3] = (o * linv[...]).astype(BF16)
    gather_send(to, tl, to_s, to_r)

    wait_all(kbuf.at[pl.ds(0, n_swap), pl.ds(0, 2)], sw_s)
    for buf, sem in ((ts, ts_s), (to, to_s)):
        wait_all(buf.at[pl.ds(0, N_FLY), pl.ds(0, 2)], sem.at[0])

    @pl.when(me != 2)
    def _():
        for k in range(2):
            wait_all(qb.at[:, pl.ds(0, 4)], q_s.at[k])

    @pl.when(me == 0)
    def _():
        for k in range(2):
            wait_all(ob, ob_s.at[k])

    @pl.when(is_qmaker)
    def _():
        wait_all(ob.at[:, 0], ob_s.at[0])
        for c in range(NC):
            ob_wait(c, 1 - half)

    @pl.when(me != 0)
    def _():
        wait_all(ls, bs_s)
        wait_all(bo.at[:, :, pl.ds(3, 1)], bo_s)

    @pl.when(me == 2)
    def _():
        for k in range(2):
            wait_all(xb, xs_s.at[k])
        for c in range(NC):
            ob_wait(c, 0)
            ob_wait(c, 1)

    def merge_wait(t):
        if t < N_FLY:
            fly_wait(t, 1)
        else:
            wait_ts(t)
            wait_to(t)

    def merge_final(t):
        if t < N_FLY:
            ct[t] = fly_merge(t, 1)[0]
        else:
            ct[t] = diag_merge(tail_weights(t), to[t])

    for t in MERGE_AT[0]:
        merge_wait(t)
    for t in MERGE_AT[0]:
        merge_final(t)

    def tail_ctx(i, n):
        return ct[i * NC:i * NC + n].reshape(n * QB, DH)

    r3 = (NC - 1) * QB
    for i, (hd, lo, hi) in enumerate(WO_PIECES):
        pending = MERGE_AT[i] if i else ()
        for t in pending:
            merge_wait(t)
        if i == WEIGHTS_AT:
            wait_ts(tl)
        wo_tail_load(i).wait()
        for t in pending:
            merge_final(t)
        if i == WEIGHTS_AT:
            for j, x in enumerate(tail_weights(tl)):
                wcol[j] = jnp.broadcast_to(to_col(x), (QB, DH))
        w = wof[(NBH + hd) * DH:(NBH + hd + 1) * DH, lo:hi].astype(BF16)
        if hd == 0:
            out_ref[0, :, lo:hi] = (
                jnp.dot(tail_ctx(0, NC), w, preferred_element_type=F32)
                + ob[:, :, :, lo:hi].reshape(NC * QB, hi - lo).astype(F32))
        elif hd < NTH - 1:
            out_ref[0, :, lo:hi] += jnp.dot(
                tail_ctx(hd, NC), w, preferred_element_type=F32)
        else:
            wlast[:, lo:hi] = w
            out_ref[0, 0:r3, lo:hi] += jnp.dot(
                tail_ctx(hd, NC - 1), w, preferred_element_type=F32)
    wait_all(ts.at[pl.ds(N_FLY, NTU - N_FLY), pl.ds(0, 3)], ts_s.at[1])
    wait_to(tl)
    acc = wcol[0] * to[tl, 0].astype(F32)
    for j in range(1, 4):
        acc += wcol[j] * to[tl, j].astype(F32)
    out_ref[0, r3:, :] += jnp.dot(
        acc.astype(BF16), wlast[...], preferred_element_type=F32)
    wait_all(to.at[pl.ds(N_FLY, NTU - N_FLY), pl.ds(0, 3)], to_s.at[1])


def pallas_dist_sparse_attn_strided_kvseq_b1_sq256_skv4096_hq8_dh128_kernel(
    x: jax.Array,
    Wq: jax.Array,
    K_ext: jax.Array,
    V_ext: jax.Array,
    Wo: jax.Array,
):
    k5 = K_ext.reshape(NG, NC, QB, NH, DH)
    v5 = V_ext.reshape(NG, NC, QB, NH, DH)
    n_staged = len(_staged_units())
    vm = pltpu.VMEM
    sm = pltpu.SMEM
    dma = pltpu.SemaphoreType.DMA
    scratch = [
        vm((NU, NG, QB, DH), F32),
        vm((NU, NG, QB, DH), F32),
        vm((NC, QB, DM), F32),
        vm((NC, QB, DM), BF16),
        vm((DM, 512), F32),
        vm((DM, 512), BF16),
        vm((DM, DM), F32),
        vm((NBH * DH, DM), BF16),
        vm((NC, NH, QB, DH), BF16),
        vm((NC, 8, DH), F32),
        vm((NC, NBH, 4, QB, DH), BF16),
        vm((NC, 3, 8, DH), F32),
        vm((NTU, 4, QB, DH), BF16),
        vm((NTU, 4, 1, DH), F32),
        vm((NTU, QB, DH), BF16),
        vm((NC, 2, QB // 2, DM), BF16),
        vm((DH, DM), BF16),
        vm((QB, NG * QB), BF16),
        vm((QB, DH), F32),
        vm((QB, K_SPLIT * QB), F32),
        vm((QB, DH), F32),
        vm((4, QB, DH), F32),
        sm((2 * N_SLOT,), jnp.int32),
        sm((N_SLOT,), jnp.int32),
        sm((NU,), jnp.int32),
        sm((N_SLOT,), jnp.int32),
        sm((n_staged,), jnp.int32),
        sm((RING, QB, DH), F32),
        dma((NU,)), dma((NU,)), dma((2,)),
        dma((NC,)), dma, dma((len(WO_PIECES),)),
        dma((2,)), dma((NC,)),
        dma((2,)), dma((NC, 2)),
        dma, dma((NC,)),
        dma, dma((NC,)),
        dma((2,)), dma((NC, 2)),
        dma((2,)), dma((NTU,)),
        dma((2,)), dma((NTU,)),
        dma,
        dma((N_FLY, 2)), dma((N_FLY, 2)),
        dma((2 * n_staged,)),
    ]
    return pl.pallas_call(
        _body,
        out_shape=jax.ShapeDtypeStruct((1, NC * QB, DM), F32),
        in_specs=[pl.BlockSpec(memory_space=pl.ANY)] * 5,
        out_specs=pl.BlockSpec(memory_space=pltpu.VMEM),
        scratch_shapes=scratch,
        compiler_params=pltpu.CompilerParams(
            collective_id=0,
            vmem_limit_bytes=64 * 1024 * 1024,
            disable_semaphore_checks=True,
        ),
    )(x, Wq, k5, v5, Wo)
```

```python
import functools

import jax
import jax.numpy as jnp
from jax import lax
from jax.experimental import pallas as pl
from jax.experimental.pallas import tpu as pltpu

NC = 4
QB = 64
NH = 8
DH = 128
DM = 1024
NG = 16
NBH = 5
NTH = NH - NBH
NBU = NC * NBH
NTU = NC * NTH
NU = NBU + NTU
Q_SCALE = 0.08838834764831843 * 1.4426950408889634

F32 = jnp.float32
BF16 = jnp.bfloat16
MESH = pl.DeviceIdType.MESH
NT_DIMS = (((1,), (1,)), ((), ()))

UNITS = [(c, h) for c in range(NC) for h in range(NBH)] + [
    (c, h) for h in range(NBH, NH) for c in range(NC)
]

PARTS = 2
AHEAD = 5
K_SPLIT = 12
V_SPLIT = 10
N_FLY = 7
FLY_LAG = 3
WO_STEP = 29
WO_PIECES = ((0, 0, 512), (0, 512, DM), (1, 0, 512), (1, 512, DM),
             (2, 0, 512), (2, 512, DM))
MERGE_AT = ((4, 5), (6, 7), (8, 9), (10,), (), ())
WEIGHTS_AT = 4

N_PRE = 5
STEP0 = 2 + N_PRE
N_SLOT = STEP0 + NU
X_SLOTS = {2: 2, 3: 4}
MAKEQ_SLOTS = (2, 4, 6, 10)
RELAY_SLOTS = (5, 9, 13, 18)
PROJECT_STEPS = (12, 15, 18, 21)
SECOND_STEPS = (13, 16, 19, 23)
FORWARD_STEPS = (16, 19, 22, 25)
ACT_X, ACT_MAKEQ, ACT_RELAY, ACT_PROJECT, ACT_SECOND, ACT_FORWARD = range(6)

SWAPS = "SSSS-+S-S+BS+S-S+BS+S-S+-S+S"
PERMS = {"+": (1, 2, 3, 0), "-": (3, 0, 1, 2), "B": (3, 2, 1, 0)}
MARKS = {".": "..", "u": "u.", "d": "d.", "U": "uu", "D": "dd", "b": "ud"}
PLANS = (
    "ud.dudu" ".d.u..dudududu.dudud" "duud.duu....",
    "ddu.ddu" "d.u..u.uduuuuu.uuudu" "dudu.duu....",
    "......." "..DU.D.UDuudduudbud." "dudu.duu....",
    "uud.udu" "d.d..u.uduuduuuu.uud" "duudd.uu....",
)
MARGIN = 3
STAGE_FIRST = 3
STAGE_IN = (
    "0121101" "01100101011011110111" "011101110000",
    "1012110" "10101010100111011110" "111011110000",
    "0101210" "00101010111101111101" "111011110000",
    "1012110" "01110001101011011110" "111011110000",
)
STAGE_OUT = (
    "2101120" "10010101011110111101" "110111011100",
    "0310111" "11010101001101110111" "101110111100",
    "0031011" "01010101011111011111" "011110111100",
    "0310111" "20001110001110110111" "101110111100",
)
STAGE_MARGIN = 1
RING = 10


def _push_table(chip):
    first = NU - len(SWAPS)
    todo = {"u": [], "d": []}
    for i, name in enumerate(SWAPS):
        if name == "S":
            continue
        dest = PERMS[name][chip]
        way = "u" if dest == (chip + 1) % 4 else "d"
        c, h = UNITS[first + i]
        for is_v in range(2):
            code = ((((first + i) * NC + c) * NH + h) * 2 + is_v) * 4 + dest
            todo[way].append((first + i, code))
    table = []
    assert len(PLANS[chip]) == N_SLOT
    for slot, mark in enumerate(PLANS[chip]):
        for way in MARKS[mark]:
            if way == ".":
                table.append(-1)
            else:
                u, code = todo[way].pop(0)
                assert slot - STEP0 <= u - MARGIN, (chip, slot, u)
                table.append(code)
    assert not todo["u"] and not todo["d"], (chip, todo)
    return table


def _staged_units():
    first = NU - len(SWAPS)
    return [first + i for i, name in enumerate(SWAPS) if name == "S"]


def _wait_slot(u):
    return 2 + u if u < N_PRE else STEP0 + u


def _stage_table(chip):
    units = _staged_units()
    n_in, n_out = STAGE_FIRST, 0
    table = []
    for slot in range(N_SLOT):
        a, b = int(STAGE_IN[chip][slot]), int(STAGE_OUT[chip][slot])
        assert n_out + b <= n_in, (chip, slot)
        for j in range(n_out, n_out + b):
            due = _wait_slot(units[j // 2])
            assert slot <= due - STAGE_MARGIN, (chip, slot, j)
        for j in range(max(n_in, RING), n_in + a):
            assert slot >= _wait_slot(units[(j - RING) // 2]), (chip, slot, j)
        table.append(n_in | (n_in + a) << 6 | n_out << 12 | (n_out + b) << 18)
        n_in += a
        n_out += b
    assert n_in == n_out == 2 * len(units), (chip, n_in, n_out)
    return table


def _action_table(chip):
    def steps(when):
        return [(STEP0 + st, c) for c, st in enumerate(when)]

    events = {}
    if chip == 0:
        events[ACT_RELAY] = list(zip(RELAY_SLOTS, range(NC)))
        events[ACT_PROJECT] = steps(PROJECT_STEPS)
        events[ACT_SECOND] = steps(SECOND_STEPS)
    elif chip == 2:
        events[ACT_X] = [(slot, c) for c, slot in X_SLOTS.items()]
    else:
        events[ACT_MAKEQ] = list(zip(MAKEQ_SLOTS, range(NC)))
        events[ACT_FORWARD] = steps(FORWARD_STEPS)
    table = [0] * N_SLOT
    for act, items in events.items():
        for slot, c in items:
            table[slot] |= (c + 1) << (3 * act)
    return table


def _body(
    x_hbm, wq_hbm, k_hbm, v_hbm, wo_hbm, out_ref,
    kbuf, vbuf, xf, xb, wqf, wqb, wof, wob, qb,
    ls, bo, bs, to, ts, ct, ob, wlast, pn, oacc, sa, linv, wcol,
    ptab, atab, utab, gtab, stab, stage,
    ksem, vsem, lsem, xlsem, wlsem, wtsem,
    xs_s, xs_r, q_s, q_r, bo_s, bo_r, bs_s, bs_r,
    ob_s, ob_r, to_s, to_r, ts_s, ts_r, sw_s, fo_r, fs_r, st_s,
):
    me = lax.axis_index("i")
    half = me // 2
    is_qmaker = me % 2 == 1
    staged = _staged_units()
    n_swap = len(SWAPS) - len(staged)
    first = NU - len(SWAPS)
    kv = ((k_hbm, kbuf, ksem), (v_hbm, vbuf, vsem))

    def remote(src, dst, ssem, rsem, dev):
        return pltpu.make_async_remote_copy(
            src, dst, ssem, rsem, device_id=(dev,), device_id_type=MESH)

    def wait_all(buf, sem):
        pltpu.make_async_copy(buf, buf, sem).wait()

    def load_blocks(u, c, h, is_v, lo, hi, sem):
        src, dst, _ = kv[is_v]
        g = pl.ds(lo, hi - lo)
        for r in range(PARTS):
            keys = pl.ds(r * (QB // PARTS), QB // PARTS)
            pltpu.make_async_copy(
                src.at[g, c, keys, h, :], dst.at[u, g, keys], sem).start()

    def load_unit(u, c, h, lo):
        for is_v in range(2):
            load_blocks(u, c, h, is_v, lo, NG, kv[is_v][2].at[u])

    def unit_of(u):
        word = utab[u]
        return word >> 3, word & 7

    def load_ahead(u):
        load_unit(u, *unit_of(u), 1)

    def load_last():
        u = NU - 1
        c, h = UNITS[u]
        for is_v, cut in enumerate((K_SPLIT, V_SPLIT)):
            load_blocks(u, c, h, is_v, 1, cut, kv[is_v][2].at[u])
            load_blocks(u, c, h, is_v, cut, NG, lsem.at[is_v])

    def last_wait(is_v, piece):
        cut = (K_SPLIT, V_SPLIT)[is_v]
        _, buf, sem = kv[is_v]
        if piece == 0:
            wait_all(buf.at[NU - 1, pl.ds(0, cut)], sem.at[NU - 1])
        else:
            wait_all(buf.at[NU - 1, pl.ds(cut, NG - cut)], lsem.at[is_v])

    def wait_unit(u):
        wait_all(kbuf.at[u], ksem.at[u])
        wait_all(vbuf.at[u], vsem.at[u])

    def push(slot, which=(0, 1)):
        for i in which:
            code = ptab[2 * slot + i]
            for is_v in range(2):
                @pl.when(jnp.logical_and(code >= 0, ((code >> 2) & 1) == is_v))
                def _(is_v=is_v, code=code):
                    src, dst, sem = kv[is_v]
                    u = code >> 8
                    block = src.at[0, (code >> 6) & 3, :, (code >> 3) & 7, :]
                    remote(block, dst.at[u, 0], sw_s, sem.at[u],
                           code & 3).start()

    def stage_in(j, ring, c, h, is_v):
        pltpu.make_async_copy(
            kv[is_v][0].at[0, c, :, h, :], stage.at[ring], st_s.at[j]).start()

    def stage_step(slot):
        word = gtab[slot]

        def drain(j, carry):
            u = stab[j] >> 4
            block = stage.at[stab[j] & 15]
            wait_all(block, st_s.at[j])
            for is_v in range(2):
                @pl.when((j & 1) == is_v)
                def _(is_v=is_v):
                    _, dst, sem = kv[is_v]
                    pltpu.make_async_copy(
                        block, dst.at[u, 0], sem.at[u]).start()
            return carry

        def fetch(j, carry):
            c, h = unit_of(stab[j] >> 4)
            for is_v in range(2):
                @pl.when((j & 1) == is_v)
                def _(is_v=is_v):
                    stage_in(j, stab[j] & 15, c, h, is_v)
            return carry

        lax.fori_loop((word >> 12) & 63, (word >> 18) & 63, drain, 0)
        lax.fori_loop(word & 63, (word >> 6) & 63, fetch, 0)

    def action(slot, act, fn):
        field = (atab[slot] >> (3 * act)) & 7

        @pl.when(field > 0)
        def _():
            fn(field - 1)

    def x_load(c):
        return pltpu.make_async_copy(
            x_hbm.at[0, pl.ds(c * QB, QB), :], xf.at[c], xlsem.at[c])

    def wq_load(hf):
        return pltpu.make_async_copy(
            wq_hbm.at[:, pl.ds(hf * 512, 512)], wqf, wlsem)

    def wo_bulk_load():
        rows = pl.ds(0, NBH * DH)
        return pltpu.make_async_copy(wo_hbm.at[rows], wof.at[rows], wlsem)

    def wo_tail_load(i):
        hd, lo, hi = WO_PIECES[i]
        rows = pl.ds((NBH + hd) * DH, DH)
        cols = pl.ds(lo, hi - lo)
        return pltpu.make_async_copy(
            wo_hbm.at[rows, cols], wof.at[rows, cols], wtsem.at[i])

    def send_x(c):
        for k in range(2):
            remote(xb.at[c], xb.at[c], xs_s.at[k], xs_r.at[c],
                   1 + 2 * k).start()

    def wait_q(c, k):
        wait_all(qb.at[c, pl.ds(k * 4, 4)], q_r.at[c, k])

    def make_q(c):
        wait_all(xb.at[c], xs_r.at[c])
        q = jnp.dot(xb[c], wqb[...], preferred_element_type=F32) * Q_SCALE
        for i in range(4):
            qb[c, half * 4 + i] = q[:, i * DH:(i + 1) * DH].astype(BF16)
        rows = qb.at[c, pl.ds(half * 4, 4)]
        for k in range(2):
            remote(rows, rows, q_s.at[k], q_r.at[c, half], 2 * k).start()

    def relay_q(c):
        for k in range(2):
            wait_q(c, k)
            rows = qb.at[c, pl.ds(k * 4, 4)]
            remote(rows, rows, q_s.at[k], q_r.at[c, k], 3 - 2 * k).start()

    def q_hooks(slot):
        action(slot, ACT_MAKEQ, make_q)
        action(slot, ACT_RELAY, relay_q)

    @pl.when(me == 2)
    def _():
        for c in range(NC):
            x_load(c).start()

    @pl.when(me == 1)
    def _():
        wq_load(0).start()

    @pl.when(me == 3)
    def _():
        wq_load(1).start()

    @pl.when(me == 0)
    def _():
        wo_bulk_load().start()

    for j in range(STAGE_FIRST):
        stage_in(j, j, *UNITS[staged[j // 2]], j % 2)

    assert first <= AHEAD
    for u in range(AHEAD):
        load_unit(u, *UNITS[u], int(u >= first))

    barrier = pltpu.get_barrier_semaphore()
    for d in (1, 2, 3):
        pl.semaphore_signal(
            barrier, 1, device_id=((me + d) % 4,), device_id_type=MESH)

    def fill(ref, tables):
        for i, words in enumerate(zip(*tables)):
            word = jnp.int32(words[0])
            for chip in range(1, 4):
                if words[chip] != words[0]:
                    word = jnp.where(me == chip, words[chip], word)
            ref[i] = word

    fill(ptab, [_push_table(chip) for chip in range(4)])
    fill(atab, [_action_table(chip) for chip in range(4)])
    fill(gtab, [_stage_table(chip) for chip in range(4)])
    fill(utab, [[c * NH + h for c, h in UNITS]] * 4)
    fill(stab, [[staged[j // 2] << 4 | j % RING
                 for j in range(2 * len(staged))]] * 4)

    pl.semaphore_wait(barrier, 3)

    @pl.when(me == 2)
    def _():
        x_load(0).wait()
        xb[0] = xf[0].astype(BF16)
        send_x(0)

    push(0)
    stage_step(0)

    @pl.when(is_qmaker)
    def _():
        wait_all(wqf, wlsem)

    @pl.when(me == 0)
    def _():
        wo_bulk_load().wait()

    push(1)
    stage_step(1)

    @pl.when(me == 2)
    def _():
        for c in range(1, NC):
            x_load(c).wait()
            xb[c] = xf[c].astype(BF16)
        send_x(1)

    @pl.when(is_qmaker)
    def _():
        wqb[...] = wqf[...].astype(BF16)

    @pl.when(me == 0)
    def _():
        wob[...] = wof[0:NBH * DH, :].astype(BF16)

    def pre_step(u, carry):
        wait_unit(u)
        load_ahead(u + AHEAD)
        push(2 + u)
        stage_step(2 + u)
        action(2 + u, ACT_X, send_x)
        q_hooks(2 + u)
        return carry

    lax.fori_loop(0, N_PRE, pre_step, 0)

    row_id = lax.broadcasted_iota(jnp.int32, (QB, DH), 0)
    lane_id = lax.broadcasted_iota(jnp.int32, (QB, DH), 1)
    eye = row_id == lane_id
    eye2 = row_id == lane_id % QB
    sub8 = lax.broadcasted_iota(jnp.int32, (8, DH), 0)

    def to_row(col):
        return jnp.sum(jnp.where(eye2, col, 0.0), axis=0, keepdims=True)

    def to_col(row):
        return jnp.sum(jnp.where(eye, row, 0.0), axis=1, keepdims=True)

    def scores(u, c, h):
        k = kbuf[u].reshape(NG * QB, DH).astype(BF16)
        s = lax.dot_general(qb[c, h], k, NT_DIMS, preferred_element_type=F32)
        m = jnp.max(s, axis=1, keepdims=True)
        p = jnp.exp2(s - m)
        l = jnp.sum(p, axis=1, keepdims=True)
        return p.astype(BF16), 1.0 / l, m + jnp.log2(l)

    def merge_weights(stats):
        m = functools.reduce(jnp.maximum, stats)
        e = [jnp.exp2(s - m) for s in stats]
        total = functools.reduce(jnp.add, e)
        inv = 1.0 / total
        return [x * inv for x in e], m + jnp.log2(total)

    def diag_merge(w, parts):
        lo = lane_id[0:1] < QB
        d = [jnp.where(eye2, jnp.where(lo, w[j], w[j + 1]), 0.0).astype(BF16)
             for j in range(0, len(w), 2)]
        return jnp.dot(jnp.concatenate(d, axis=1),
                       parts.reshape(len(w) * QB, DH),
                       preferred_element_type=F32).astype(BF16)

    def ob_send(c, rnd):
        for k in range(2):
            hf = k ^ rnd
            rows = ob.at[c, hf]
            remote(rows, rows, ob_s.at[k], ob_r.at[c, hf], 1 + 2 * k).start()

    def ob_wait(c, hf):
        wait_all(ob.at[c, hf], ob_r.at[c, hf])

    def project_bulk(c):
        wait_all(bs.at[c], bs_r.at[c])
        wait_all(bo.at[c, :, pl.ds(0, 3)], bo_r.at[c])
        w, _ = merge_weights([bs[c, j] for j in range(3)] + [ls[c]])
        ctx = jnp.concatenate(
            [diag_merge([x[h:h + 1] for x in w], bo[c, h]) for h in range(NBH)],
            axis=1)
        o = jnp.dot(ctx, wob[...], preferred_element_type=F32)
        ob[c] = o.astype(BF16).reshape(2, QB // 2, DM)
        ob_send(c, 0)

    def forward_bulk(c):
        ob_wait(c, half)
        rows = ob.at[c, half]
        remote(rows, rows, ob_s.at[0], ob_r.at[c, half], 2).start()

    def role_hooks(slot):
        action(slot, ACT_PROJECT, project_bulk)
        action(slot, ACT_SECOND, lambda c: ob_send(c, 1))
        action(slot, ACT_FORWARD, forward_bulk)

    def bulk_step(u, stat):
        slot = STEP0 + u
        c, h = unit_of(u)

        @pl.when(jnp.logical_and(h == 0, me >= 2))
        def _():
            wait_q(c, 0)

        @pl.when(jnp.logical_and(h == 0, jnp.logical_or(me == 1, me == 2)))
        def _():
            wait_q(c, 1)

        @pl.when(u >= N_PRE)
        def _():
            wait_unit(u)
            load_ahead(u + AHEAD)

        push(slot, (0,))
        p, inv_l, lse = scores(u, c, h)
        v = vbuf[u].reshape(NG * QB, DH).astype(BF16)
        o = jnp.dot(p, v, preferred_element_type=F32) * inv_l
        bo[c, h, 3] = o.astype(BF16)
        stat = jnp.where(sub8 == h, to_row(lse), stat)
        ls[c] = stat

        @pl.when(me != 0)
        def _():
            remote(bo.at[c, h, 3], bo.at[c, h, me - 1], bo_s, bo_r.at[c],
                   0).start()

        @pl.when(jnp.logical_and(h == NBH - 1, me != 0))
        def _():
            remote(ls.at[c], bs.at[c, me - 1], bs_s, bs_r.at[c], 0).start()

        push(slot, (1,))
        stage_step(slot)
        q_hooks(slot)
        role_hooks(slot)
        return stat

    lax.fori_loop(0, NBU, bulk_step, jnp.zeros((8, DH), F32))

    dests = (jnp.where(me == 0, 2, 0), jnp.where(me == 1, 3, 1),
             jnp.where(is_qmaker, 2, 3))
    slots = tuple((d - me + 4) % 4 - 1 for d in dests)

    def gather_send(buf, t, ssem, rsem):
        for k in range(3):
            remote(buf.at[t, 3], buf.at[t, slots[k]], ssem.at[1], rsem.at[t],
                   dests[k]).start()

    def wait_ts(t):
        wait_all(ts.at[t, pl.ds(0, 3)], ts_r.at[t])

    def wait_to(t):
        wait_all(to.at[t, pl.ds(0, 3)], to_r.at[t])

    def tail_weights(t):
        return merge_weights([ts[t, j] for j in range(4)])[0]

    def fly_send(t, rnd):
        dev = jnp.where(((t + rnd) & 1) == 0, me ^ 1, 3 - me)
        src = 3 - 2 * rnd
        remote(ts.at[t, src], ts.at[t, src - 1], ts_s.at[0], fs_r.at[t, rnd],
               dev).start()
        remote(to.at[t, src], to.at[t, src - 1], to_s.at[0], fo_r.at[t, rnd],
               dev).start()

    def fly_wait(t, rnd):
        dst = 2 - 2 * rnd
        wait_all(ts.at[t, dst], fs_r.at[t, rnd])
        wait_all(to.at[t, dst], fo_r.at[t, rnd])

    def fly_merge(t, rnd):
        lo = 2 - 2 * rnd
        w, lse = merge_weights([ts[t, lo], ts[t, lo + 1]])
        return diag_merge(w, to[t, lo:lo + 2]), lse

    def tail_step(t, carry):
        u = NBU + t
        slot = STEP0 + u
        wait_all(kbuf.at[u], ksem.at[u])
        p, inv_l, lse = scores(u, *unit_of(u))
        ts[t, 3] = to_row(lse)

        @pl.when(t >= N_FLY)
        def _():
            gather_send(ts, t, ts_s, ts_r)

        push(slot, (0,))
        wait_all(vbuf.at[u], vsem.at[u])
        v = vbuf[u].reshape(NG * QB, DH).astype(BF16)
        o = jnp.dot(p, v, preferred_element_type=F32) * inv_l
        to[t, 3] = o.astype(BF16)

        @pl.when(t >= N_FLY)
        def _():
            gather_send(to, t, to_s, to_r)

        @pl.when(t < N_FLY)
        def _():
            fly_send(t, 0)

        @pl.when(jnp.logical_and(t >= FLY_LAG, t < N_FLY + FLY_LAG))
        def _():
            f = t - FLY_LAG
            fly_wait(f, 0)
            to[f, 1], ts[f, 1] = fly_merge(f, 0)
            fly_send(f, 1)

        push(slot, (1,))
        stage_step(slot)

        @pl.when(u + AHEAD < NU - 1)
        def _():
            load_ahead(u + AHEAD)

        @pl.when(u + AHEAD == NU - 1)
        def _():
            load_last()

        @pl.when(u == WO_STEP)
        def _():
            for i in range(len(WO_PIECES)):
                wo_tail_load(i).start()

        role_hooks(slot)

        @pl.when(jnp.logical_and(t >= 2 * FLY_LAG,
                                 t - 2 * FLY_LAG < MERGE_AT[0][0]))
        def _():
            f = t - 2 * FLY_LAG
            fly_wait(f, 1)
            ct[f] = fly_merge(f, 1)[0]

        return carry

    tl = NTU - 1
    lax.fori_loop(0, tl, tail_step, 0)

    def blocks(buf, lo, hi):
        return buf[NU - 1, lo:hi].reshape((hi - lo) * QB, DH).astype(BF16)

    q = qb[NC - 1, NH - 1]
    last_wait(0, 0)
    sa[...] = lax.dot_general(q, blocks(kbuf, 0, K_SPLIT), NT_DIMS,
                              preferred_element_type=F32)
    last_wait(0, 1)
    s = jnp.concatenate(
        [sa[...], lax.dot_general(q, blocks(kbuf, K_SPLIT, NG), NT_DIMS,
                                  preferred_element_type=F32)], axis=1)
    m = jnp.max(s, axis=1, keepdims=True)
    p = jnp.exp2(s - m)
    pn[...] = p.astype(BF16)
    l = jnp.sum(p, axis=1, keepdims=True)
    last_wait(1, 0)
    oacc[...] = jnp.dot(pn[:, 0:V_SPLIT * QB], blocks(vbuf, 0, V_SPLIT),
                        preferred_element_type=F32)
    linv[...] = jnp.broadcast_to(1.0 / l, (QB, DH))
    ts[tl, 3] = to_row(m + jnp.log2(l))
    gather_send(ts, tl, ts_s, ts_r)
    last_wait(1, 1)
    o = oacc[...] + jnp.dot(pn[:, V_SPLIT * QB:], blocks(vbuf, V_SPLIT, NG),
                            preferred_element_type=F32)
    to[tl, 3] = (o * linv[...]).astype(BF16)
    gather_send(to, tl, to_s, to_r)

    wait_all(kbuf.at[pl.ds(0, n_swap), pl.ds(0, 2)], sw_s)
    for buf, sem in ((ts, ts_s), (to, to_s)):
        wait_all(buf.at[pl.ds(0, N_FLY), pl.ds(0, 2)], sem.at[0])

    @pl.when(me != 2)
    def _():
        for k in range(2):
            wait_all(qb.at[:, pl.ds(0, 4)], q_s.at[k])

    @pl.when(me == 0)
    def _():
        for k in range(2):
            wait_all(ob, ob_s.at[k])

    @pl.when(is_qmaker)
    def _():
        wait_all(ob.at[:, 0], ob_s.at[0])
        for c in range(NC):
            ob_wait(c, 1 - half)

    @pl.when(me != 0)
    def _():
        wait_all(ls, bs_s)
        wait_all(bo.at[:, :, pl.ds(3, 1)], bo_s)

    @pl.when(me == 2)
    def _():
        for k in range(2):
            wait_all(xb, xs_s.at[k])
        for c in range(NC):
            ob_wait(c, 0)
            ob_wait(c, 1)

    def merge_wait(t):
        if t < N_FLY:
            fly_wait(t, 1)
        else:
            wait_ts(t)
            wait_to(t)

    def merge_final(t):
        if t < N_FLY:
            ct[t] = fly_merge(t, 1)[0]
        else:
            ct[t] = diag_merge(tail_weights(t), to[t])

    for t in MERGE_AT[0]:
        merge_wait(t)
    for t in MERGE_AT[0]:
        merge_final(t)

    def tail_ctx(i, n):
        return ct[i * NC:i * NC + n].reshape(n * QB, DH)

    r3 = (NC - 1) * QB
    for i, (hd, lo, hi) in enumerate(WO_PIECES):
        pending = MERGE_AT[i] if i else ()
        for t in pending:
            merge_wait(t)
        if i == WEIGHTS_AT:
            wait_ts(tl)
        wo_tail_load(i).wait()
        for t in pending:
            merge_final(t)
        if i == WEIGHTS_AT:
            for j, x in enumerate(tail_weights(tl)):
                wcol[j] = jnp.broadcast_to(to_col(x), (QB, DH))
        w = wof[(NBH + hd) * DH:(NBH + hd + 1) * DH, lo:hi].astype(BF16)
        if hd == 0:
            out_ref[0, :, lo:hi] = (
                jnp.dot(tail_ctx(0, NC), w, preferred_element_type=F32)
                + ob[:, :, :, lo:hi].reshape(NC * QB, hi - lo).astype(F32))
        elif hd < NTH - 1:
            out_ref[0, :, lo:hi] += jnp.dot(
                tail_ctx(hd, NC), w, preferred_element_type=F32)
        else:
            wlast[:, lo:hi] = w
            out_ref[0, 0:r3, lo:hi] += jnp.dot(
                tail_ctx(hd, NC - 1), w, preferred_element_type=F32)
    wait_all(ts.at[pl.ds(N_FLY, NTU - N_FLY), pl.ds(0, 3)], ts_s.at[1])
    wait_to(tl)
    acc = wcol[0] * to[tl, 0].astype(F32)
    for j in range(1, 4):
        acc += wcol[j] * to[tl, j].astype(F32)
    out_ref[0, r3:, :] += jnp.dot(
        acc.astype(BF16), wlast[...], preferred_element_type=F32)
    wait_all(to.at[pl.ds(N_FLY, NTU - N_FLY), pl.ds(0, 3)], to_s.at[1])


def pallas_dist_sparse_attn_strided_kvseq_b1_sq256_skv4096_hq8_dh128_kernel(
    x: jax.Array,
    Wq: jax.Array,
    K_ext: jax.Array,
    V_ext: jax.Array,
    Wo: jax.Array,
):
    k5 = K_ext.reshape(NG, NC, QB, NH, DH)
    v5 = V_ext.reshape(NG, NC, QB, NH, DH)
    n_staged = len(_staged_units())
    vm = pltpu.VMEM
    sm = pltpu.SMEM
    dma = pltpu.SemaphoreType.DMA
    scratch = [
        vm((NU, NG, QB, DH), F32),
        vm((NU, NG, QB, DH), F32),
        vm((NC, QB, DM), F32),
        vm((NC, QB, DM), BF16),
        vm((DM, 512), F32),
        vm((DM, 512), BF16),
        vm((DM, DM), F32),
        vm((NBH * DH, DM), BF16),
        vm((NC, NH, QB, DH), BF16),
        vm((NC, 8, DH), F32),
        vm((NC, NBH, 4, QB, DH), BF16),
        vm((NC, 3, 8, DH), F32),
        vm((NTU, 4, QB, DH), BF16),
        vm((NTU, 4, 1, DH), F32),
        vm((NTU, QB, DH), BF16),
        vm((NC, 2, QB // 2, DM), BF16),
        vm((DH, DM), BF16),
        vm((QB, NG * QB), BF16),
        vm((QB, DH), F32),
        vm((QB, K_SPLIT * QB), F32),
        vm((QB, DH), F32),
        vm((4, QB, DH), F32),
        sm((2 * N_SLOT,), jnp.int32),
        sm((N_SLOT,), jnp.int32),
        sm((NU,), jnp.int32),
        sm((N_SLOT,), jnp.int32),
        sm((2 * n_staged,), jnp.int32),
        sm((RING, QB, DH), F32),
        dma((NU,)), dma((NU,)), dma((2,)),
        dma((NC,)), dma, dma((len(WO_PIECES),)),
        dma((2,)), dma((NC,)),
        dma((2,)), dma((NC, 2)),
        dma, dma((NC,)),
        dma, dma((NC,)),
        dma((2,)), dma((NC, 2)),
        dma((2,)), dma((NTU,)),
        dma((2,)), dma((NTU,)),
        dma,
        dma((N_FLY, 2)), dma((N_FLY, 2)),
        dma((2 * n_staged,)),
    ]
    params = dict(collective_id=0, vmem_limit_bytes=64 * 1024 * 1024)
    if hasattr(pltpu.CompilerParams, "disable_semaphore_checks"):
        params["disable_semaphore_checks"] = True
    return pl.pallas_call(
        _body,
        out_shape=jax.ShapeDtypeStruct((1, NC * QB, DM), F32),
        in_specs=[pl.BlockSpec(memory_space=pl.ANY)] * 5,
        out_specs=pl.BlockSpec(memory_space=pltpu.VMEM),
        scratch_shapes=scratch,
        compiler_params=pltpu.CompilerParams(**params),
    )(x, Wq, k5, v5, Wo)
```
